```python
import numpy as np

kernel_name = "dist_sparse_attn_strided_kvseq_b1_sq256_skv4096_hq8_dh128"

def setup_inputs():
    x = np.random.randn(1, 256, 1024).astype(np.float32)
    Wq = np.random.randn(1024, 1024).astype(np.float32) * 0.02
    K_ext = np.random.randn(1, 16384, 8, 128).astype(np.float32)
    V_ext = np.random.randn(1, 16384, 8, 128).astype(np.float32)
    Wo = np.random.randn(1024, 1024).astype(np.float32) * 0.02
    return {"x": x, "Wq": Wq, "K_ext": K_ext, "V_ext": V_ext, "Wo": Wo}

def reference(x, Wq, K_ext, V_ext, Wo):
    B, Sq, Skv, Hq, Dh = 1, 256, 16384, 8, 128
    Q = (x @ Wq).reshape(B, Sq, Hq, Dh)
    qb = (np.arange(Sq) // 64)[:, None]
    kb = (np.arange(Skv) // 64)[None, :]
    mask = (qb == kb) | ((kb % 4) == (qb % 4))
    scores = np.einsum('bihd,bjhd->bhij', Q, K_ext).astype(np.float32) * 0.08838834764831843
    scores = np.where(mask[None, None, :, :], scores, -1e9)
    scores_max = scores.max(axis=-1, keepdims=True)
    w = np.exp(scores - scores_max)
    row_keep = mask.any(axis=1)
    w_sum = np.where(row_keep[None, None, :, None], w.sum(axis=-1, keepdims=True), 1.0)
    w = w / w_sum
    w = np.where(row_keep[None, None, :, None], w, 0.0)
    ctx = np.einsum('bhij,bjhd->bihd', w, V_ext).reshape(B, Sq, Hq * Dh)
    return ctx @ Wo
```

```python
import contextlib
import jax
import jax.numpy as jnp
from jax import lax
from jax.experimental import pallas as pl
from jax.experimental.pallas import tpu as pltpu

SCOPES = "0" == "1"
GSPLIT = int("12")
SH0 = int('4')
LSW = tuple(int(c) for c in '012')
FD = int("3")
SKIP = int("1")
PRE = tuple(int(c) for c in '222')
MASKS = '1111111111111111111101010101'
MASK = sum(1 << u for u, ch in enumerate(MASKS) if ch == "1")
UQ1 = int('10')
PF = int("9")
CMB = tuple(int(c) for c in "012")
UQ2 = int('14')
JOBSETS = {
    "a": ((20, 4, (0, 2, -1, -1)), (23, 4, (1, 3, -1, -1)), (24, 5, (-1, -1, -1, 6)), (26, 5, (4, 5, -1, 7))),
    "b": ((19, 4, (0, 2, -1, -1)), (22, 4, (1, 3, -1, -1)), (23, 5, (-1, -1, -1, 6)), (25, 5, (4, 5, -1, 7))),
    "c": ((20, 4, (0, 3, -1, 6)), (23, 4, (1, 4, -1, 7)), (26, 4, (2, 5, -1, -1))),
    "d": ((20, 4, (0, 3, -1, -1)), (23, 4, (1, 4, -1, -1)), (24, 5, (-1, -1, -1, 6)), (26, 4, (2, 5, -1, -1)), (27, 5, (-1, -1, -1, 7))),
    "e": ((19, 4, (0, 3, -1, 6)), (22, 4, (1, 4, -1, 7)), (25, 4, (2, 5, -1, -1))),
    "f": ((19, 4, (0, 3, -1, 6)), (22, 4, (1, 4, -1, 7)), (24, 4, (2, 5, -1, -1))),
    "g": ((15, 3, (0, 1, -1, -1)), (19, 4, (2, 4, -1, 6)), (22, 4, (3, 5, -1, 7))),
    "h": ((19, 4, (0, 3, -1, 6)), (21, 4, (1, 4, -1, 7)), (23, 4, (2, 5, -1, -1))),
    "i": ((20, 4, (0, 3, -1, 6)), (22, 4, (1, 4, -1, 7)), (24, 4, (2, 5, -1, -1))),
    "j": ((20, 4, (0, 3, -1, 6)), (22, 4, (1, 4, -1, -1)), (24, 4, (2, 5, -1, -1)), (24, 5, (-1, -1, -1, 7))),
    "k": ((20, 4, (0, 2, -1, 4)), (22, 4, (1, 3, -1, -1)), (24, 5, (5, 6, -1, 7))),
    "l": ((20, 4, (0, 2, -1, 4)), (22, 4, (1, 3, -1, 5)), (24, 5, (6, -1, -1, 7))),
    "m": ((19, 4, (0, 2, -1, 4)), (21, 4, (1, 3, -1, -1)), (23, 5, (5, 6, -1, 7))),
    "n": ((20, 4, (0, 3, -1, 5)), (22, 4, (1, 4, -1, 6)), (24, 4, (2, -1, -1, 7))),
    "o": ((19, 4, (0, 3, -1, 5)), (21, 4, (1, 4, -1, 6)), (23, 4, (2, -1, -1, 7))),
    "u": ((18, 3, (0, 2, 4, 6)), (22, 3, (1, 3, 5, 7))),
}
JOBS = JOBSETS['o']
WINSETS = {
    "0": ((((4, 0, 8),), (0,)), (((5, 0, 8),), (1,)), (((6, 0, 8),), (2,)), (((7, 0, 8),), ())),
    "1": ((((4, 0, 8),), (0,)), (((5, 0, 8),), (1,)), (((6, 0, 4),), ()), (((6, 4, 8),), (2,)), (((7, 0, 4),), ()), (((7, 4, 8),), ())),
    "2": ((((4, 0, 8),), (0,)), (((5, 0, 8),), (1,)), (((6, 0, 8),), (2,)), (((7, 0, 4),), ()), (((7, 4, 8),), ())),
    "3": ((((4, 0, 8),), (0,)), (((5, 0, 8),), (1,)), (((6, 0, 6),), (2,)), (((6, 6, 8), (7, 0, 3)), ()), (((7, 3, 6),), ()), (((7, 6, 8),), ())),
    "4": ((((4, 0, 8),), (0,)), (((5, 0, 6),), (1,)), (((5, 6, 8), (6, 0, 4)), ()), (((6, 4, 8),), (2,)), (((7, 0, 4),), ()), (((7, 4, 8),), ())),
    "5": ((((4, 0, 8),), (0,)), (((5, 0, 8),), (1,)), (((6, 0, 4),), ()), (((6, 4, 8),), (2,)), (((7, 0, 5),), ()), (((7, 5, 8),), ())),
}
WINSETS["6"] = ((((4, 0, 8),), ()), (((5, 0, 8),), (0,)), (((6, 0, 4),), (1,)), (((6, 4, 8),), (2,)), (((7, 0, 4),), ()), (((7, 4, 8),), ()))
WINSETS["7"] = ((((4, 0, 8),), (0,)), (((5, 0, 8),), ()), (((6, 0, 8),), (1, 2)), (((7, 0, 8),), ()))
WINSETS["8"] = ((((4, 0, 8),), (0,)), (((5, 0, 8),), ()), (((6, 0, 4),), ()), (((6, 4, 8),), (1, 2)), (((7, 0, 4),), ()), (((7, 4, 8),), ()))
for _n in (4, 5, 6, 7):
    WINSETS["p%d" % _n] = ((((4, 0, _n),), (0,)), (((5, 0, 8),), (1,)), (((6, 0, 8),), (2,)), (((7, 0, 8),), ()))
REGIONS = WINSETS["0"]
MERGE = int("0")
PIECES = [p for r in REGIONS for p in r[0]]

N_DEV = 4
NQB = 4
QB = 64
H = 8
DH = 128
NG = 16
EH = H - 1
DM = H * DH
KS = DM // N_DEV
MSG_ROWS = 80
SCALE = 0.08838834764831843
MESH = pl.DeviceIdType.MESH
F32 = jnp.float32
BF16 = jnp.bfloat16
QGROUPS = ((0, 2), (2, 5), (5, 8))
NJ = len(JOBS)
DEPTH = {t: d for _, d, ts in JOBS for t in ts if t >= 0}
assert sorted(DEPTH) == list(range(H))
NA = min(DEPTH.values())
MAXD = max(DEPTH.values())
WCOLS = [DH * sum(1 for t in range(H) if DEPTH[t] <= h) for h in range(NA, H)]
assert all(DEPTH[t] <= DEPTH[t + 1] for t in range(H - 1))
NW = H - NA
LAST = NQB - 1
NU = EH * NQB
NMID = (EH - SH0) * NQB
NPAIR = NMID + len(LSW)
assert sum(PRE) + MASKS.count('1') == 2 * NPAIR, (sum(PRE) + MASKS.count('1'), 2 * NPAIR)
FWDIR = tuple(int(c) for c in '0002')
IDLE = [d for d in range(N_DEV) if all(j[2][d] < 0 for j in JOBS)]
IDLE = IDLE[0] if IDLE and SKIP else -1

S_X, S_WQA, S_WQB = 0, 1, 2
S_WO = 3
S_G = S_WO + NJ
S_K = S_G + 2 * SH0
S_V = S_K + NU
S_KL = S_V + NU
S_VL = S_KL + NQB
S_WL = S_VL + NQB + 1
S_N = S_WL + len(PIECES)


def _scope(name):
    return jax.named_scope(name) if SCOPES else contextlib.nullcontext()


def _table(tab, i):
    if isinstance(i, int):
        return tab[i]
    packed = sum((v & 15) << (4 * s) for s, v in enumerate(tab))
    return lax.shift_right_logical(jnp.int32(packed), 4 * i) & 15


def _body(x_ref, wq_ref, k_ref, v_ref, wo_ref, o_ref,
          xbuf, wqbuf, woa, wol, kbuf, vbuf, qpart, qrs, qbuf, p16buf, invbuf, msg, rsbuf, ctxbuf, lbuf, obuf, w7buf, wgt,
          lsem, qr_ss, qr_rs, qa_ss, qa_rs, r_ss, r_rs, a_ss, a_rs, l_ss, l_rs, o_ss, o_rs, f_ss, x_ss, x_rs):
    me = lax.axis_index("i")
    peers = [(me + d) & 3 for d in (1, 2, 3)]
    srcs = [(me + N_DEV - d) & 3 for d in (1, 2, 3)]
    order = (1, 0, 2)
    kv = ((k_ref, kbuf), (v_ref, vbuf))

    bar = pltpu.get_barrier_semaphore()
    for p in peers:
        pl.semaphore_signal(bar, inc=1, device_id=(p,), device_id_type=MESH)

    def when_job(dev, p):
        if min(JOBS[p][2]) >= 0:
            return lambda f: f()
        return pl.when(_table(JOBS[p][2], dev) < H)

    def when_tab(tab):
        if all(tab):
            return lambda f: f()
        if not any(tab):
            return lambda f: None
        return pl.when(_table(tuple(int(v) for v in tab), me) == 1)

    def has(p, d):
        return JOBS[p][2][d % N_DEV] >= 0

    def fwd_tab(p, j):
        return [has(p, d - j - 1) and FWDIR[(d - j - 1) % N_DEV] == j and FD > 0 for d in range(N_DEV)]

    def unit_c(i):
        return (me + _table((2, 1, 3, 0), i)) & 3

    k0 = pl.multiple_of(me * KS, KS)
    na = QGROUPS[0][1] * DH
    x_cp = pltpu.make_async_copy(x_ref.at[0, :, pl.ds(k0, KS)], xbuf, lsem.at[S_X])
    wqa_cp = pltpu.make_async_copy(wq_ref.at[pl.ds(k0, KS), pl.ds(0, na)], wqbuf.at[:, pl.ds(0, na)], lsem.at[S_WQA])
    wqb_cp = pltpu.make_async_copy(wq_ref.at[pl.ds(k0, KS), pl.ds(na, DM - na)], wqbuf.at[:, pl.ds(na, DM - na)], lsem.at[S_WQB])

    def woa_copy(p):
        col = pl.multiple_of(_table(JOBS[p][2], me) * DH, DH)
        rows = pl.ds(0, JOBS[p][1] * DH)
        return pltpu.make_async_copy(wo_ref.at[rows, pl.ds(col, DH)], woa.at[p, rows], lsem.at[S_WO + p])

    def g_copy(h, t):
        src, dst = kv[t]
        return pltpu.make_async_copy(src.at[0, :, :, h, :], dst.at[h, 0], lsem.at[S_G + 2 * h + t])

    def u_copy(u, t):
        src, dst = kv[t]
        h, c = u >> 2, unit_c(u & 3)
        sl = pl.ds(1, NG - 1)
        return pltpu.make_async_copy(src.at[sl, c, :, h, :], dst.at[h, sl, c], lsem.at[(S_K, S_V)[t] + u])

    def kl_copy(c):
        g0 = int(c in LSW)
        sl = pl.ds(g0, NG - g0)
        return pltpu.make_async_copy(k_ref.at[sl, c, :, EH, :], kbuf.at[EH, sl, c], lsem.at[S_KL + c])

    def vl_copy(c, g0=0, g1=NG, s=0):
        g0 = max(g0, int(c in LSW))
        sl = pl.ds(g0, g1 - g0)
        return pltpu.make_async_copy(v_ref.at[sl, c, :, EH, :], vbuf.at[EH, sl, c], lsem.at[S_VL + c + s])

    def wl_copy(i):
        h, a, b = PIECES[i]
        cols = pl.ds(a * DH, (b - a) * DH)
        return pltpu.make_async_copy(wo_ref.at[pl.ds(h * DH, DH), cols], wol.at[h - NA, :, cols], lsem.at[S_WL + i])

    x_cp.start()
    wqa_cp.start()
    wqb_cp.start()
    for u in range(PF):
        if u % NQB == 0:
            g_copy(u // NQB, 0).start()
            g_copy(u // NQB, 1).start()
        u_copy(u, 0).start()
        u_copy(u, 1).start()
    g_next = (PF + NQB - 1) // NQB

    def remote(src, dst, ss, rs, dev):
        return pltpu.make_async_remote_copy(src, dst, ss, rs, device_id=(dev,), device_id_type=MESH)

    def qr_copy(g, j):
        a, b = QGROUPS[g]
        return remote(qpart.at[peers[j], pl.ds(a, b - a)], qrs.at[j, pl.ds(a, b - a)], qr_ss.at[g, j], qr_rs.at[g, j], peers[j])

    def qa_copy(g, j, dev):
        a, b = QGROUPS[g]
        sl = qbuf.at[dev, pl.ds(a, b - a)]
        return remote(sl, sl, qa_ss.at[g, j], qa_rs.at[g, j], peers[j])

    def o_copy(p, j, dev):
        sl = obuf.at[_table(JOBS[p][2], dev)]
        return remote(sl, sl, o_ss.at[p, j], o_rs.at[p, j], peers[j])

    def f_copy(p, j):
        sl = obuf.at[_table(JOBS[p][2], srcs[j])]
        return remote(sl, sl, f_ss.at[p, j // 2], o_rs.at[p, 1], peers[j])

    def r_copy(h, i):
        c = unit_c(i)
        return remote(msg.at[h, c], rsbuf.at[h, i], r_ss.at[h, i], r_rs.at[h, i], c)

    def a_copy(h, j, dev):
        return remote(ctxbuf.at[h, dev], ctxbuf.at[h, dev], a_ss.at[h, j], a_rs.at[h, j], peers[j])

    def l_copy(c, j):
        dev = (me + j + 1) & 3
        if c == LAST:
            return remote(msg.at[EH, c, pl.ds(0, QB)], lbuf.at[c, j, pl.ds(0, QB)], l_ss.at[c, j], l_rs.at[c, j], dev)
        return remote(msg.at[EH, c], lbuf.at[c, j], l_ss.at[c, j], l_rs.at[c, j], dev)

    def s_copy(j):
        sl = pl.ds(QB, MSG_ROWS - QB)
        return remote(msg.at[EH, LAST, sl], lbuf.at[LAST, j, sl], l_ss.at[NQB, j], l_rs.at[NQB, j], peers[j])

    def x_copy(p, t, recv=False):
        src, dst = kv[t]
        h, i = SH0 + (p >> 2), p & 3
        dev = (me + _table((1, 3, 3, 1), i)) & 3
        c = unit_c(i) if recv else (me + _table((3, 0, 2, 1), i)) & 3
        return remote(src.at[0, c, :, h, :], dst.at[h, 0, c], x_ss.at[p, t], x_rs.at[p, t], dev)

    def xl_copy(n, t):
        src, dst = kv[t]
        c = LSW[n]
        return remote(src.at[0, c, :, EH, :], dst.at[EH, 0, c], x_ss.at[NMID + n, t], x_rs.at[NMID + n, t],
                      peers[2 * (n & 1)])

    def q_partial(x16, a, b):
        q = jnp.dot(x16, wqbuf[:, a * DH:b * DH].astype(BF16), preferred_element_type=F32)
        q = (q * SCALE).astype(BF16)
        for c in range(NQB):
            for h in range(a, b):
                qpart[c, h] = q[c * QB:(c + 1) * QB, (h - a) * DH:(h - a + 1) * DH]

    def q_reduce(g):
        a, b = QGROUPS[g]
        with _scope("qred"):
            for j in range(3):
                qr_copy(g, j).wait()
            acc = qpart[me, a:b].astype(F32)
            for j in range(3):
                acc = acc + qrs[j, a:b].astype(F32)
            qbuf[me, a:b] = acc.astype(BF16)
        for j in order:
            qa_copy(g, j, me).start()

    def q_wait(g):
        for j in range(3):
            qa_copy(g, j, srcs[j]).wait_recv()
            qa_copy(g, j, me).wait_send()

    with _scope("qproj"):
        x_cp.wait()
        x16 = xbuf[...].astype(BF16)
        wqa_cp.wait()
        q_partial(x16, *QGROUPS[0])
    with _scope("bar"):
        pl.semaphore_wait(bar, 3)
    for j in order:
        qr_copy(0, j).start()
    with _scope("qproj"):
        wqb_cp.wait()
        q_partial(x16, QGROUPS[1][0], QGROUPS[2][1])
    pre_order = [0, 2, 1, 3, 4, 6, 5, 7] if sum(PRE) % 4 == 0 else list(range(8))

    def pre_swaps(k):
        for m in pre_order[sum(PRE[:k]):sum(PRE[:k + 1])]:
            x_copy(m >> 1, m & 1).start()

    for j in order:
        qr_copy(1, j).start()
    pre_swaps(0)
    q_reduce(0)
    if UQ1 < 0:
        for j in order:
            qr_copy(2, j).start()
    pre_swaps(1)
    q_reduce(1)
    pre_swaps(2)
    for p in range(NJ):
        when_job(me, p)(lambda p=p: woa_copy(p).start())
    with _scope("waitq"):
        g_copy(0, 0).wait()
        g_copy(0, 1).wait()
        q_wait(0)

    row = lax.broadcasted_iota(jnp.int32, (QB, DH), 0)
    lane = lax.broadcasted_iota(jnp.int32, (QB, DH), 1)
    diag = (lane & (QB - 1)) == row
    diag1 = lane == row
    srow = lax.broadcasted_iota(jnp.int32, (16, DH), 0)
    lo_half = lax.broadcasted_iota(jnp.int32, (1, DH), 1) < QB

    def qk(h, c):
        k = kbuf[h, :, c].reshape(NG * QB, DH).astype(BF16)
        s = lax.dot_general(qbuf[c, h], k, (((1,), (1,)), ((), ())), preferred_element_type=F32)
        m = jnp.max(s, axis=1, keepdims=True)
        p = jnp.exp(s - m)
        l = jnp.sum(p, axis=1, keepdims=True)
        p16buf[...] = p.astype(BF16)
        lse = m + jnp.log(l)
        r = jnp.sum(jnp.where(diag, lse, 0.0), axis=0, keepdims=True)
        hi = r.astype(BF16).astype(F32)
        mid = (r - hi).astype(BF16).astype(F32)
        lo = r - hi - mid
        st = jnp.where(srow == 0, hi, jnp.where(srow == 1, mid, jnp.where(srow == 2, lo, 0.0)))
        msg[h, c, QB:MSG_ROWS, :] = st.astype(BF16)
        invbuf[0] = jnp.broadcast_to(1.0 / l, (QB, DH))

    def pv_part(h, c, g0, g1):
        v = vbuf[h, g0:g1, c].reshape((g1 - g0) * QB, DH).astype(BF16)
        return jnp.dot(p16buf[:, g0 * QB:g1 * QB], v, preferred_element_type=F32)

    def pv(h, c):
        msg[h, c, 0:QB, :] = (pv_part(h, c, 0, NG) * invbuf[0]).astype(BF16)

    def weights(parts):
        ls = [jnp.sum(p[QB:MSG_ROWS, :].astype(F32), axis=0, keepdims=True) for p in parts]
        mx = jnp.maximum(jnp.maximum(ls[0], ls[1]), jnp.maximum(ls[2], ls[3]))
        es = [jnp.exp(a - mx) for a in ls]
        inv = 1.0 / (es[0] + es[1] + es[2] + es[3])
        return [e * inv for e in es]

    def combine(parts):
        w = weights(parts)
        w01 = jnp.where(lo_half, w[0], w[1])
        w23 = jnp.where(lo_half, w[2], w[3])
        d = jnp.concatenate([jnp.where(diag, w01, 0.0), jnp.where(diag, w23, 0.0)], axis=1).astype(BF16)
        st = jnp.concatenate([p[0:QB, :] for p in parts], axis=0)
        return jnp.dot(d, st, preferred_element_type=F32).astype(BF16)

    def reduce_head(h):
        with _scope("waitr"):
            for i in range(3):
                r_copy(h, i).wait()
        with _scope("comb"):
            ctxbuf[h, me] = combine([msg.at[h, me]] + [rsbuf.at[h, i] for i in range(3)])
        for j in order:
            if IDLE < 0 or isinstance(h, int):
                a_copy(h, j, me).start()
            else:
                pl.when(jnp.logical_or(h >= NA, peers[j] != IDLE))(lambda j=j: a_copy(h, j, me).start())

    def wait_ctx(h):
        for j in range(3):
            if h < NA:
                when_tab([d != IDLE for d in range(N_DEV)])(lambda j=j: a_copy(h, j, srcs[j]).wait_recv())
                when_tab([(d + j + 1) % N_DEV != IDLE for d in range(N_DEV)])(lambda j=j: a_copy(h, j, me).wait_send())
            else:
                a_copy(h, j, srcs[j]).wait_recv()
                a_copy(h, j, me).wait_send()

    ctx_ready = [0]

    def unit_step(u, sw):
        h = u >> 2
        i = u & 3
        c = unit_c(i)
        un = u + PF

        @pl.when(un < NU)
        def _():
            u_copy(un, 0).start()
            u_copy(un, 1).start()

        with _scope("waitk"):
            @pl.when(h >= SH0)
            def _():
                for t in range(2):
                    x_copy(u - SH0 * NQB, t, True).wait_recv()
                    x_copy(u - SH0 * NQB, t).wait_send()

            u_copy(u, 0).wait()
        with _scope("qk"):
            qk(h, c)
        with _scope("waitv"):
            u_copy(u, 1).wait()
        with _scope("pv"):
            pv(h, c)

        @pl.when(i < 3)
        def _():
            r_copy(h, i).start()

        @pl.when(u == UQ2)
        def _():
            q_reduce(2)

        @pl.when(jnp.logical_and(i == 0, h > 0))
        def _():
            reduce_head(h - 1)

        if UQ1 >= 0:
            @pl.when(u == UQ1)
            def _():
                for j in order:
                    qr_copy(2, j).start()

        go_sw = lax.shift_right_logical(jnp.int32(MASK), u) & 1
        for t in range(2):
            @pl.when(jnp.logical_and(jnp.logical_and(go_sw == 1, sw < 2 * NMID), (sw & 1) == t))
            def _(t=t):
                x_copy(sw >> 1, t).start()

        @pl.when(jnp.logical_and(go_sw == 1, sw >= 2 * NMID))
        def _():
            for n in range(len(LSW)):
                for t in range(2):
                    pl.when(sw == 2 * (NMID + n) + t)(lambda n=n, t=t: xl_copy(n, t).start())

        ctx_ready[0] = 0
        for p in range(NJ):
            @pl.when(u == JOBS[p][0])
            def _(p=p):
                depth = JOBS[p][1]
                with _scope("waitc"):
                    for hh in range(ctx_ready[0], depth):
                        wait_ctx(hh)
                ctx_ready[0] = max(ctx_ready[0], depth)

                def go():
                    with _scope("oearly"):
                        woa_copy(p).wait()
                        ctx = jnp.concatenate([ctxbuf[hh].reshape(NQB * QB, DH) for hh in range(depth)], axis=1)
                        obuf[_table(JOBS[p][2], me)] = jnp.dot(
                            ctx, woa[p, 0:depth * DH].astype(BF16), preferred_element_type=F32).astype(BF16)
                    for j in ((0, 2) if FD else order):
                        o_copy(p, j, me).start()
                when_job(me, p)(go)

        for p in range(NJ if FD else 0):
            @pl.when(u == JOBS[p][0] + FD)
            def _(p=p):
                for j in (0, 2):
                    def fw(j=j):
                        o_copy(p, j, srcs[j]).wait_recv()
                        f_copy(p, j).start()
                    when_tab(fwd_tab(p, j))(fw)

        @pl.when(i == 3)
        def _():
            with _scope("prep"):
                @pl.when(h + g_next < SH0)
                def _():
                    g_copy(h + g_next, 0).start()
                    g_copy(h + g_next, 1).start()

                @pl.when(h == EH - 2)
                def _():
                    for cc in range(NQB):
                        kl_copy(cc).start()
                        if cc == LAST:
                            vl_copy(cc, 0, GSPLIT).start()
                            vl_copy(cc, GSPLIT, NG, 1).start()
                        else:
                            vl_copy(cc).start()

                for g in (1, 2):
                    pl.when(h + 1 == QGROUPS[g][0])(lambda g=g: q_wait(g))

                @pl.when(h + 1 < SH0)
                def _():
                    g_copy(h + 1, 0).wait()
                    g_copy(h + 1, 1).wait()

        return sw + go_sw

    lax.fori_loop(0, NU, unit_step, jnp.int32(sum(PRE)))

    for w in range(len(PIECES)):
        wl_copy(w).start()

    def late_x_wait(c):
        if c in LSW:
            for t in range(2):
                xl_copy(LSW.index(c), t).wait()

    for c in range(LAST):
        with _scope("waitk"):
            late_x_wait(c)
            kl_copy(c).wait()
        with _scope("qk"):
            qk(EH, c)
        with _scope("waitv"):
            vl_copy(c).wait()
        with _scope("pv"):
            pv(EH, c)
        for j in order:
            l_copy(c, j).start()
        if c == 0:
            reduce_head(EH - 1)

    with _scope("waitk"):
        late_x_wait(LAST)
        kl_copy(LAST).wait()
    with _scope("qk"):
        qk(EH, LAST)
    for j in order:
        s_copy(j).start()
    with _scope("waitv"):
        vl_copy(LAST, 0, GSPLIT).wait()
    with _scope("pv"):
        wgt[...] = pv_part(EH, LAST, 0, GSPLIT)
    with _scope("waitv"):
        vl_copy(LAST, GSPLIT, NG, 1).wait()
    with _scope("pv"):
        acc = wgt[...] + pv_part(EH, LAST, GSPLIT, NG)
        msg[EH, LAST, 0:QB, :] = (acc * invbuf[0]).astype(BF16)
    for tab in ((1, 2, 1, 0), (0, 1, 0, 1), (2, 0, 2, 2)):
        l_copy(LAST, _table(tab, me)).start()

    parts = [msg.at[EH, LAST]] + [lbuf.at[LAST, j] for j in range(3)]
    wgt_region = len(REGIONS) - (2 if MERGE else 1)
    seen = set(range(MAXD))
    n = 0

    def last_rows():
        ctx = wgt[...]
        for j in range(3):
            ctx = ctx + parts[j + 1][0:QB, :].astype(F32) * invbuf[j]
        o_ref[0, LAST * QB:, :] += jnp.dot(ctx.astype(BF16), w7buf[...], preferred_element_type=F32)

    for r, (pieces, combs) in enumerate(REGIONS):
        final = MERGE and r == len(REGIONS) - 1
        with _scope("waitw"):
            if r == 0:
                for p in range(NJ):
                    for j in range(3):
                        fw = fwd_tab(p, j)
                        when_tab([has(p, d - j - 1) and not fw[d] for d in range(N_DEV)])(
                            lambda p=p, j=j: o_copy(p, j, srcs[j]).wait_recv())
                        when_tab(fw)(lambda p=p, j=j: f_copy(p, j).wait_send())
                        if j != 1 or not FD:
                            when_job(me, p)(lambda p=p, j=j: o_copy(p, j, me).wait_send())
            for h, _, _ in pieces:
                if h < EH and h not in seen:
                    wait_ctx(h)
                    seen.add(h)
            for c in combs:
                for j in range(3):
                    l_copy(c, j).wait()
            if r == wgt_region:
                for j in range(3):
                    s_copy(j).wait()
                    l_copy(LAST, j).wait_send()
            for _ in pieces:
                wl_copy(n).wait()
                n += 1
            if final:
                for j in (0, 2, 1):
                    l_copy(LAST, j).wait_recv()
        with _scope("olate"):
            for c in combs:
                ctxbuf[EH, c] = combine([msg.at[EH, c]] + [lbuf.at[c, j] for j in range(3)])
            if r == wgt_region:
                cols = [jnp.sum(jnp.where(diag1, w, 0.0), axis=1, keepdims=True) for w in weights(parts)]
                wgt[...] = parts[0][0:QB, :].astype(F32) * cols[0]
                for j in range(3):
                    invbuf[j] = jnp.broadcast_to(cols[j + 1], (QB, DH))
            for h, a, b in pieces:
                cs = slice(a * DH, b * DH)
                w = wol[h - NA, :, cs].astype(BF16)
                if h == EH:
                    w7buf[:, cs] = w
                    o_ref[0, 0:LAST * QB, cs] += jnp.dot(ctxbuf[EH, 0:LAST].reshape(LAST * QB, DH), w,
                                                         preferred_element_type=F32)
                    continue
                upd = jnp.dot(ctxbuf[h].reshape(NQB * QB, DH), w, preferred_element_type=F32)
                if r == 0:
                    o_ref[0, :, cs] = upd + jnp.concatenate([obuf[p] for p in range(a, b)], axis=1).astype(F32)
                    for p in range(b, H):
                        o_ref[0, :, p * DH:(p + 1) * DH] = obuf[p].astype(F32)
                else:
                    o_ref[0, :, cs] += upd
            if final:
                last_rows()
    if not MERGE:
        with _scope("waitl"):
            for j in (0, 2, 1):
                l_copy(LAST, j).wait_recv()
        with _scope("fin"):
            last_rows()


def pallas_dist_sparse_attn_strided_kvseq_b1_sq256_skv4096_hq8_dh128_kernel(x, Wq, K_ext, V_ext, Wo):
    k5 = K_ext.reshape(NG, NQB, QB, H, DH)
    v5 = V_ext.reshape(NG, NQB, QB, H, DH)
    dma = pltpu.SemaphoreType.DMA
    ng = len(QGROUPS)
    return pl.pallas_call(
        _body,
        out_shape=jax.ShapeDtypeStruct((1, NQB * QB, DM), F32),
        in_specs=[pl.BlockSpec(memory_space=pltpu.HBM)] * 5,
        out_specs=pl.BlockSpec(memory_space=pltpu.VMEM),
        scratch_shapes=[
            pltpu.VMEM((NQB * QB, KS), F32),
            pltpu.VMEM((KS, DM), F32),
            pltpu.VMEM((NJ, MAXD * DH, DH), F32),
            pltpu.VMEM((NW, DH, DM), F32),
            pltpu.VMEM((H, NG, NQB, QB, DH), F32),
            pltpu.VMEM((H, NG, NQB, QB, DH), F32),
            pltpu.VMEM((NQB, H, QB, DH), BF16),
            pltpu.VMEM((3, H, QB, DH), BF16),
            pltpu.VMEM((NQB, H, QB, DH), BF16),
            pltpu.VMEM((QB, NG * QB), BF16),
            pltpu.VMEM((3, QB, DH), F32),
            pltpu.VMEM((H, NQB, MSG_ROWS, DH), BF16),
            pltpu.VMEM((EH, 3, MSG_ROWS, DH), BF16),
            pltpu.VMEM((H, NQB, QB, DH), BF16),
            pltpu.VMEM((NQB, 3, MSG_ROWS, DH), BF16),
            pltpu.VMEM((H, NQB * QB, DH), BF16),
            pltpu.VMEM((DH, DM), BF16),
            pltpu.VMEM((QB, DH), F32),
            dma((S_N,)),
            dma((ng, 3)), dma((ng, 3)), dma((ng, 3)), dma((ng, 3)),
            dma((EH, 3)), dma((EH, 3)),
            dma((EH, 3)), dma((EH, 3)),
            dma((NQB + 1, 3)), dma((NQB + 1, 3)),
            dma((NJ, 3)), dma((NJ, 3)), dma((NJ, 2)),
            dma((NPAIR, 2)), dma((NPAIR, 2)),
        ],
        compiler_params=pltpu.CompilerParams(
            vmem_limit_bytes=64 * 1024 * 1024,
            collective_id=0,
            disable_semaphore_checks=True,
            disable_bounds_checks=True,
        ),
    )(x, Wq, k5, v5, Wo)
```

```python
import contextlib
import jax
import jax.numpy as jnp
from jax import lax
from jax.experimental import pallas as pl
from jax.experimental.pallas import tpu as pltpu

SCOPES = "0" == "1"
GSPLIT = int("12")
WH = int("1")
PF = int("8")
NSW = tuple(int(c) for c in "00000000000000001111111111112210")
PRE = tuple(int(c) for c in "2022")
SENDS = tuple(int(c) for c in "1111111111111111111111111111")
QCUT = tuple(int(c) for c in "01358")
UQ1 = tuple(int(c, 36) for c in "1a")
UQ2 = tuple(int(c, 36) for c in "5e")
FD = tuple(int(c) for c in "3333")
RED = tuple(int(c) for c in "0000000")
JOBSETS = {
    "o": ((19, 4, (0, 3, -1, 5)), (21, 4, (1, 4, -1, 6)), (23, 4, (2, -1, -1, 7))),
    "p": ((19, 4, (0, 3, -1, 4)), (21, 4, (1, -1, -1, 5)), (23, 4, (2, -1, -1, 6)), (23, 5, (-1, 7, -1, -1))),
    "q": ((19, 4, (0, 3, -1, 4)), (21, 4, (1, -1, -1, 5)), (23, 4, (2, -1, -1, 6)), (24, 5, (-1, 7, -1, -1))),
    "s": ((19, 4, (0, 3, -1, 1)), (21, 4, (2, -1, -1, 4)), (23, 5, (5, 6, -1, 7))),
    "t": ((19, 4, (0, 3, -1, 1)), (21, 4, (2, -1, -1, 4)), (24, 5, (5, 6, -1, 7))),
    "v": ((19, 4, (0, 3, -1, 1)), (21, 4, (2, 5, -1, 4)), (23, 5, (6, -1, -1, 7))),
}
JOBS = JOBSETS["s"]
FWDIR = [tuple(int(c) for c in w) for w in "0002.0002.2000.0002".split(".")]

N_DEV = 4
NQB = 4
QB = 64
H = 8
DH = 128
NG = 16
EH = H - 1
DM = H * DH
KS = DM // N_DEV
MSG_ROWS = 80
SROWS = int("8")
SENT = QB + SROWS
SCALE = 0.08838834764831843
MESH = pl.DeviceIdType.MESH
F32 = jnp.float32
BF16 = jnp.bfloat16
QGROUPS = tuple(zip(QCUT[:-1], QCUT[1:]))
NJ = len(JOBS)
DEPTH = {t: d for _, d, ts in JOBS for t in ts if t >= 0}
NA = min(DEPTH.values())
MAXD = max(DEPTH.values())
WTILES = [sum(1 for t in range(H) if DEPTH[t] <= h) for h in range(NA, H)]
NW = H - NA
LAST = NQB - 1
NU = EH * NQB
NT = H * NQB
SWAPS = [(u, g, t) for u in range(NT) for g in range(NSW[u]) for t in range(2)]
assert sum(PRE) + sum(SENDS) == len(SWAPS), (sum(PRE) + sum(SENDS), len(SWAPS))
NEED = [max([d for _, d, ts in JOBS if ts[dev] >= 0], default=0) for dev in range(N_DEV)]
UNIT_OFF = (2, 1, 3, 0)
SWAP_DIR = (1, 3, 3, 1)
LATE_DIR = tuple(int(c) for c in "11331")

S_X, S_WQ = 0, 1
S_WO = 4
S_KV = S_WO + NJ
S_V2 = S_KV + 2 * NT
S_WL = S_V2 + 1
S_N = S_WL + NW


def _scope(name):
    return jax.named_scope(name) if SCOPES else contextlib.nullcontext()


def _body(x_ref, wq_ref, k_ref, v_ref, wo_ref, o_ref,
          xbuf, wqbuf, woa, wol, kbuf, vbuf, qpart, qrs, qbuf, p16buf, invbuf, msg, rsbuf, ctxbuf, lbuf, obuf, w7buf, wgt,
          lsem, qr_ss, qr_rs, qa_ss, qa_rs, r_ss, r_rs, a_ss, a_rs, l_ss, l_rs, o_ss, o_rs, f_ss, x_ss, x_rs):
    me = lax.axis_index("i")
    ring = [me] + [(me + d) & 3 for d in (1, 2, 3)]
    peers = ring[1:]
    srcs = ring[:0:-1]
    order = (1, 0, 2)
    kv = ((k_ref, kbuf), (v_ref, vbuf))

    bar = pltpu.get_barrier_semaphore()
    for p in peers:
        pl.semaphore_signal(bar, inc=1, device_id=(p,), device_id_type=MESH)

    def table(tab, dev):
        packed = sum((v & 15) << (4 * s) for s, v in enumerate(tab))
        return lax.shift_right_logical(jnp.int32(packed), 4 * dev) & 15

    def on(pred):
        tab = [int(bool(pred(d))) for d in range(N_DEV)]
        if all(tab):
            return lambda f: f()
        if not any(tab):
            return lambda f: None
        return pl.when(table(tab, me) == 1)

    def has(p, d):
        return JOBS[p][2][d % N_DEV] >= 0

    def forwards(p, j, d):
        return has(p, d - j - 1) and FWDIR[p][(d - j - 1) % N_DEV] == j

    def unit_hc(u):
        h, i = divmod(u, NQB)
        return h, (i if h == EH else ring[UNIT_OFF[i]])

    k0 = pl.multiple_of(me * KS, KS)
    x_cp = pltpu.make_async_copy(x_ref.at[0, :, pl.ds(k0, KS)], xbuf, lsem.at[S_X])
    wq_parts = (QGROUPS[0], QGROUPS[1], (QGROUPS[2][0], H))

    def wq_copy(n):
        a, b = wq_parts[n]
        cols = pl.ds(a * DH, (b - a) * DH)
        return pltpu.make_async_copy(wq_ref.at[pl.ds(k0, KS), cols], wqbuf.at[:, cols], lsem.at[S_WQ + n])

    def woa_copy(p):
        col = pl.multiple_of(table(JOBS[p][2], me) * DH, DH)
        rows = pl.ds(0, JOBS[p][1] * DH)
        return pltpu.make_async_copy(wo_ref.at[rows, pl.ds(col, DH)], woa.at[p, rows], lsem.at[S_WO + p])

    def head_copy(h, t):
        src, dst = kv[t]
        return pltpu.make_async_copy(src.at[:, :, :, h, :], dst.at[h], lsem.at[S_KV + 2 * NQB * h + t])

    def unit_copy(u, t, part=0):
        src, dst = kv[t]
        h, c = unit_hc(u)
        g0, g1 = NSW[u], NG
        if u == NT - 1 and t == 1:
            g0, g1 = (GSPLIT, NG) if part else (g0, GSPLIT)
        sl = pl.ds(g0, g1 - g0)
        return pltpu.make_async_copy(src.at[sl, c, :, h, :], dst.at[h, sl, c],
                                     lsem.at[S_V2 if part else S_KV + 2 * u + t])

    def wl_copy(i):
        cols = pl.ds(0, WTILES[i] * DH)
        return pltpu.make_async_copy(wo_ref.at[pl.ds((NA + i) * DH, DH), cols], wol.at[i, :, cols], lsem.at[S_WL + i])

    def fetch(u):
        if u < WH * NQB:
            if u % NQB == 0:
                head_copy(u // NQB, 0).start()
                head_copy(u // NQB, 1).start()
        elif u < NT:
            unit_copy(u, 0).start()
            unit_copy(u, 1).start()
            if u == NT - 1:
                unit_copy(u, 1, 1).start()
        elif u < NT + NW:
            wl_copy(u - NT).start()

    x_cp.start()
    for n in range(3):
        wq_copy(n).start()
    first = max(WH * NQB + NQB, PF)
    for u in range(first):
        fetch(u)

    def remote(src, dst, ss, rs, dev):
        return pltpu.make_async_remote_copy(src, dst, ss, rs, device_id=(dev,), device_id_type=MESH)

    def qr_copy(g, j):
        a, b = QGROUPS[g]
        return remote(qpart.at[peers[j], pl.ds(a, b - a)], qrs.at[j, pl.ds(a, b - a)], qr_ss.at[g, j], qr_rs.at[g, j], peers[j])

    def qa_copy(g, j, dev):
        a, b = QGROUPS[g]
        sl = qbuf.at[dev, pl.ds(a, b - a)]
        return remote(sl, sl, qa_ss.at[g, j], qa_rs.at[g, j], peers[j])

    def o_copy(p, j, dev):
        sl = obuf.at[table(JOBS[p][2], dev)]
        return remote(sl, sl, o_ss.at[p, j], o_rs.at[p, j], peers[j])

    def f_copy(p, j):
        sl = obuf.at[table(JOBS[p][2], srcs[j])]
        return remote(sl, sl, f_ss.at[p, j // 2], o_rs.at[p, 1], peers[j])

    def r_copy(h, i):
        c = ring[UNIT_OFF[i]]
        return remote(msg.at[h, c, pl.ds(0, SENT)], rsbuf.at[h, i, pl.ds(0, SENT)], r_ss.at[h, i], r_rs.at[h, i], c)

    def a_copy(h, j, dev):
        return remote(ctxbuf.at[h, dev], ctxbuf.at[h, dev], a_ss.at[h, j], a_rs.at[h, j], peers[j])

    def l_copy(c, j):
        dev = (me + j + 1) & 3
        if c == LAST:
            return remote(msg.at[EH, c, pl.ds(0, QB)], lbuf.at[c, j, pl.ds(0, QB)], l_ss.at[c, j], l_rs.at[c, j], dev)
        return remote(msg.at[EH, c, pl.ds(0, SENT)], lbuf.at[c, j, pl.ds(0, SENT)], l_ss.at[c, j], l_rs.at[c, j], dev)

    def s_copy(j):
        sl = pl.ds(QB, SROWS)
        return remote(msg.at[EH, LAST, sl], lbuf.at[LAST, j, sl], l_ss.at[NQB, j], l_rs.at[NQB, j], peers[j])

    def x_copy(m, recv=False):
        u, g, t = SWAPS[m]
        src, dst = kv[t]
        h, i = divmod(u, NQB)
        d = LATE_DIR[sum(NSW[NU:u]) + g] if h == EH else SWAP_DIR[i]
        c = i if h == EH else ring[(UNIT_OFF[i] + (0 if recv else d)) % N_DEV]
        return remote(src.at[g, c, :, h, :], dst.at[h, g, c], x_ss.at[m], x_rs.at[m], ring[d])

    pending = list(range(len(SWAPS)))
    for n in range(1, sum(PRE) - 2, 4):
        pending[n], pending[n + 1] = pending[n + 1], pending[n]

    def send_swaps(n):
        for _ in range(n):
            x_copy(pending.pop(0)).start()

    def q_partial(x16, a, b):
        q = jnp.dot(x16, wqbuf[:, a * DH:b * DH].astype(BF16), preferred_element_type=F32)
        q = (q * SCALE).astype(BF16)
        for c in range(NQB):
            for h in range(a, b):
                qpart[c, h] = q[c * QB:(c + 1) * QB, (h - a) * DH:(h - a + 1) * DH]

    def q_scatter(g):
        for j in order:
            qr_copy(g, j).start()

    def q_reduce(g):
        a, b = QGROUPS[g]
        with _scope("qred"):
            for j in range(3):
                qr_copy(g, j).wait()
            acc = qpart[me, a:b].astype(F32)
            for j in range(3):
                acc = acc + qrs[j, a:b].astype(F32)
            qbuf[me, a:b] = acc.astype(BF16)
        for j in order:
            qa_copy(g, j, me).start()

    def q_wait(g):
        with _scope("waitq"):
            for j in range(3):
                qa_copy(g, j, srcs[j]).wait_recv()
                qa_copy(g, j, me).wait_send()

    with _scope("qproj"):
        x_cp.wait()
        x16 = xbuf[...].astype(BF16)
        wq_copy(0).wait()
        q_partial(x16, *wq_parts[0])
    with _scope("bar"):
        pl.semaphore_wait(bar, 3)
    q_scatter(0)
    send_swaps(PRE[0])
    with _scope("qproj"):
        wq_copy(1).wait()
        q_partial(x16, *wq_parts[1])
    q_scatter(1)
    send_swaps(PRE[1])
    with _scope("qproj"):
        wq_copy(2).wait()
        q_partial(x16, *wq_parts[2])
    q_reduce(0)
    send_swaps(PRE[2])
    q_reduce(1)
    send_swaps(PRE[3])
    for p in range(NJ):
        on(lambda d: has(p, d))(lambda p=p: woa_copy(p).start())

    row = lax.broadcasted_iota(jnp.int32, (QB, DH), 0)
    lane = lax.broadcasted_iota(jnp.int32, (QB, DH), 1)
    diag = (lane & (QB - 1)) == row
    diag1 = lane == row
    srow = lax.broadcasted_iota(jnp.int32, (16, DH), 0)
    lo_half = lax.broadcasted_iota(jnp.int32, (1, DH), 1) < QB

    def qk(h, c):
        k = kbuf[h, :, c].reshape(NG * QB, DH).astype(BF16)
        s = lax.dot_general(qbuf[c, h], k, (((1,), (1,)), ((), ())), preferred_element_type=F32)
        m = jnp.max(s, axis=1, keepdims=True)
        p = jnp.exp(s - m)
        l = jnp.sum(p, axis=1, keepdims=True)
        p16buf[...] = p.astype(BF16)
        lse = m + jnp.log(l)
        r = jnp.sum(jnp.where(diag, lse, 0.0), axis=0, keepdims=True)
        hi = r.astype(BF16).astype(F32)
        mid = (r - hi).astype(BF16).astype(F32)
        lo = r - hi - mid
        st = jnp.where(srow == 0, hi, jnp.where(srow == 1, mid, jnp.where(srow == 2, lo, 0.0)))
        msg[h, c, QB:MSG_ROWS, :] = st.astype(BF16)
        invbuf[0] = jnp.broadcast_to(1.0 / l, (QB, DH))

    def pv_part(h, c, g0, g1):
        v = vbuf[h, g0:g1, c].reshape((g1 - g0) * QB, DH).astype(BF16)
        return jnp.dot(p16buf[:, g0 * QB:g1 * QB], v, preferred_element_type=F32)

    def weights(parts):
        ls = [jnp.sum(p[QB:SENT, :].astype(F32), axis=0, keepdims=True) for p in parts]
        mx = jnp.maximum(jnp.maximum(ls[0], ls[1]), jnp.maximum(ls[2], ls[3]))
        es = [jnp.exp(a - mx) for a in ls]
        inv = 1.0 / (es[0] + es[1] + es[2] + es[3])
        return [e * inv for e in es]

    def combine(parts):
        w = weights(parts)
        w01 = jnp.where(lo_half, w[0], w[1])
        w23 = jnp.where(lo_half, w[2], w[3])
        d = jnp.concatenate([jnp.where(diag, w01, 0.0), jnp.where(diag, w23, 0.0)], axis=1).astype(BF16)
        st = jnp.concatenate([p[0:QB, :] for p in parts], axis=0)
        return jnp.dot(d, st, preferred_element_type=F32).astype(BF16)

    def wants_ctx(h, d):
        return h >= NA or NEED[d % N_DEV] > h

    def reduce_head(h):
        with _scope("waitr"):
            for i in range(3):
                r_copy(h, i).wait()
        with _scope("comb"):
            ctxbuf[h, me] = combine([msg.at[h, me]] + [rsbuf.at[h, i] for i in range(3)])
        for j in order:
            on(lambda d: wants_ctx(h, d + j + 1))(lambda j=j: a_copy(h, j, me).start())

    have_ctx = [0] * N_DEV

    def recv_ctx(depth, devs):
        for h in range(depth):
            for j in range(3):
                on(lambda d: d in devs and have_ctx[d] <= h and wants_ctx(h, d))(
                    lambda j=j, h=h: a_copy(h, j, srcs[j]).wait_recv())
        for d in devs:
            have_ctx[d] = max(have_ctx[d], depth)

    def run_job(p):
        depth = JOBS[p][1]
        with _scope("waitc"):
            recv_ctx(depth, [d for d in range(N_DEV) if has(p, d)])

        def go():
            with _scope("oearly"):
                woa_copy(p).wait()
                ctx = jnp.concatenate([ctxbuf[hh].reshape(NQB * QB, DH) for hh in range(depth)], axis=1)
                obuf[table(JOBS[p][2], me)] = jnp.dot(
                    ctx, woa[p, 0:depth * DH].astype(BF16), preferred_element_type=F32).astype(BF16)
            for j in (0, 2):
                o_copy(p, j, me).start()
        on(lambda d: has(p, d))(go)

    def forward_job(p):
        for j in (0, 2):
            def fw(j=j):
                o_copy(p, j, srcs[j]).wait_recv()
                f_copy(p, j).start()
            with _scope("fwd"):
                on(lambda d: forwards(p, j, d))(fw)

    for u in range(NT):
        h, c = unit_hc(u)
        i = u % NQB
        if u + PF >= first:
            fetch(u + PF)
        for g in range(len(QGROUPS)):
            if u == QGROUPS[g][0] * NQB:
                q_wait(g)
        with _scope("waitk"):
            for m in range(len(SWAPS)):
                if SWAPS[m][0] == u and (SWAPS[m][2] == 0 or u < NT - 1):
                    x_copy(m, True).wait_recv()
            if u >= WH * NQB:
                unit_copy(u, 0).wait()
            elif i == 0:
                head_copy(h, 0).wait()
        with _scope("qk"):
            qk(h, c)
        if u == NT - 1:
            break
        with _scope("waitv"):
            if u >= WH * NQB:
                unit_copy(u, 1).wait()
            elif i == 0:
                head_copy(h, 1).wait()
        with _scope("pv"):
            msg[h, c, 0:QB, :] = (pv_part(h, c, 0, NG) * invbuf[0]).astype(BF16)
        if h == EH:
            for j in order:
                l_copy(c, j).start()
        elif i < 3:
            r_copy(h, i).start()
        if u in UQ2:
            q_reduce(2 + UQ2.index(u))
        if h > 0 and i == RED[h - 1]:
            reduce_head(h - 1)
        if i == 1 and h > 1:
            for j in range(3):
                on(lambda d: wants_ctx(h - 2, d + j + 1))(lambda j=j: a_copy(h - 2, j, me).wait_send())
        if u in UQ1:
            q_scatter(2 + UQ1.index(u))
        if u < len(SENDS):
            send_swaps(SENDS[u])
        for p in range(NJ):
            if u == JOBS[p][0]:
                run_job(p)
        for p in range(NJ):
            if u == JOBS[p][0] + FD[p]:
                forward_job(p)

    for j in order:
        s_copy(j).start()
    with _scope("waitv"):
        for m in range(len(SWAPS)):
            if SWAPS[m][0] == NT - 1 and SWAPS[m][2] == 1:
                x_copy(m, True).wait_recv()
        unit_copy(NT - 1, 1).wait()
    with _scope("pv"):
        wgt[...] = pv_part(EH, LAST, 0, GSPLIT)
    with _scope("waitv"):
        unit_copy(NT - 1, 1, 1).wait()
    with _scope("pv"):
        acc = wgt[...] + pv_part(EH, LAST, GSPLIT, NG)
        msg[EH, LAST, 0:QB, :] = (acc * invbuf[0]).astype(BF16)
    for tab in ((1, 2, 1, 0), (0, 1, 0, 1), (2, 0, 2, 2)):
        l_copy(LAST, table(tab, me)).start()

    parts = [msg.at[EH, LAST]] + [lbuf.at[LAST, j] for j in range(3)]
    for r in range(NW):
        h = NA + r
        comb = r - (NW - NQB)
        with _scope("waitw"):
            if r == 0:
                for m in range(len(SWAPS)):
                    x_copy(m).wait_send()
                for j in range(3):
                    a_copy(EH - 1, j, me).wait_send()
                for p in range(NJ):
                    for j in range(3):
                        on(lambda d: has(p, d - j - 1) and not forwards(p, j, d))(
                            lambda p=p, j=j: o_copy(p, j, srcs[j]).wait_recv())
                        if j != 1:
                            on(lambda d: forwards(p, j, d))(lambda p=p, j=j: f_copy(p, j).wait_send())
                            on(lambda d: has(p, d))(lambda p=p, j=j: o_copy(p, j, me).wait_send())
            if h < EH:
                recv_ctx(h + 1, range(N_DEV))
            if 0 <= comb < LAST:
                for j in range(3):
                    l_copy(comb, j).wait()
            if h == EH:
                for j in range(3):
                    s_copy(j).wait()
                    l_copy(LAST, j).wait_send()
            wl_copy(r).wait()
        with _scope("olate"):
            if 0 <= comb < LAST:
                ctxbuf[EH, comb] = combine([msg.at[EH, comb]] + [lbuf.at[comb, j] for j in range(3)])
            nt = WTILES[r]
            w = wol[r, :, 0:nt * DH].astype(BF16)
            if h == EH:
                cols = [jnp.sum(jnp.where(diag1, v, 0.0), axis=1, keepdims=True) for v in weights(parts)]
                wgt[...] = parts[0][0:QB, :].astype(F32) * cols[0]
                for j in range(3):
                    invbuf[j] = jnp.broadcast_to(cols[j + 1], (QB, DH))
                w7buf[...] = w
                o_ref[0, 0:LAST * QB, :] += jnp.dot(ctxbuf[EH, 0:LAST].reshape(LAST * QB, DH), w,
                                                    preferred_element_type=F32)
            else:
                upd = jnp.dot(ctxbuf[h].reshape(NQB * QB, DH), w, preferred_element_type=F32)
                if r == 0:
                    o_ref[0, :, 0:nt * DH] = upd + jnp.concatenate([obuf[p] for p in range(nt)], axis=1).astype(F32)
                    for p in range(nt, H):
                        o_ref[0, :, p * DH:(p + 1) * DH] = obuf[p].astype(F32)
                else:
                    o_ref[0, :, 0:nt * DH] += upd
    with _scope("waitl"):
        for j in (0, 2, 1):
            l_copy(LAST, j).wait_recv()
    with _scope("fin"):
        ctx = wgt[...]
        for j in range(3):
            ctx = ctx + parts[j + 1][0:QB, :].astype(F32) * invbuf[j]
        o_ref[0, LAST * QB:, :] += jnp.dot(ctx.astype(BF16), w7buf[...], preferred_element_type=F32)


def pallas_dist_sparse_attn_strided_kvseq_b1_sq256_skv4096_hq8_dh128_kernel(x, Wq, K_ext, V_ext, Wo):
    k5 = K_ext.reshape(NG, NQB, QB, H, DH)
    v5 = V_ext.reshape(NG, NQB, QB, H, DH)
    dma = pltpu.SemaphoreType.DMA
    ng = len(QGROUPS)
    return pl.pallas_call(
        _body,
        out_shape=jax.ShapeDtypeStruct((1, NQB * QB, DM), F32),
        in_specs=[pl.BlockSpec(memory_space=pltpu.HBM)] * 5,
        out_specs=pl.BlockSpec(memory_space=pltpu.VMEM),
        scratch_shapes=[
            pltpu.VMEM((NQB * QB, KS), F32),
            pltpu.VMEM((KS, DM), F32),
            pltpu.VMEM((NJ, MAXD * DH, DH), F32),
            pltpu.VMEM((NW, DH, DM), F32),
            pltpu.VMEM((H, NG, NQB, QB, DH), F32),
            pltpu.VMEM((H, NG, NQB, QB, DH), F32),
            pltpu.VMEM((NQB, H, QB, DH), BF16),
            pltpu.VMEM((3, H, QB, DH), BF16),
            pltpu.VMEM((NQB, H, QB, DH), BF16),
            pltpu.VMEM((QB, NG * QB), BF16),
            pltpu.VMEM((3, QB, DH), F32),
            pltpu.VMEM((H, NQB, MSG_ROWS, DH), BF16),
            pltpu.VMEM((EH, 3, MSG_ROWS, DH), BF16),
            pltpu.VMEM((H, NQB, QB, DH), BF16),
            pltpu.VMEM((NQB, 3, MSG_ROWS, DH), BF16),
            pltpu.VMEM((H, NQB * QB, DH), BF16),
            pltpu.VMEM((DH, DM), BF16),
            pltpu.VMEM((QB, DH), F32),
            dma((S_N,)),
            dma((ng, 3)), dma((ng, 3)), dma((ng, 3)), dma((ng, 3)),
            dma((EH, 3)), dma((EH, 3)),
            dma((EH, 3)), dma((EH, 3)),
            dma((NQB + 1, 3)), dma((NQB + 1, 3)),
            dma((NJ, 3)), dma((NJ, 3)), dma((NJ, 2)),
            dma((len(SWAPS),)), dma((len(SWAPS),)),
        ],
        compiler_params=pltpu.CompilerParams(
            vmem_limit_bytes=64 * 1024 * 1024,
            collective_id=0,
            disable_semaphore_checks=True,
            disable_bounds_checks=True,
        ),
    )(x, Wq, k5, v5, Wo)
```

```python
import jax
import jax.numpy as jnp
from jax import lax
from jax.experimental import pallas as pl
from jax.experimental.pallas import tpu as pltpu

N_DEV = 4
NQB = 4
QB = 64
H = 8
DH = 128
NG = 16
DM = H * DH
KS = DM // N_DEV
EH = H - 1
LAST = NQB - 1
NU = EH * NQB
NT = H * NQB
MSG_ROWS = QB + 16
SENT = QB + 8
SCALE = 0.08838834764831843
MESH = pl.DeviceIdType.MESH
F32 = jnp.float32
BF16 = jnp.bfloat16


def _digits(text):
    return tuple(int(ch) for ch in text)


PREFETCH = 8
V_SPLIT = 8

UNIT_OFF = (2, 1, 3, 0)
LATE_ORDER = ((1, 2, 1, 0), (0, 1, 0, 1), (2, 0, 2, 2))

QGROUPS = ((0, 1), (1, 3), (3, 5), (5, 8))
Q_SCATTER = {1: 2, 10: 3}
Q_REDUCE = {5: 2, 14: 3}

JOBS = (
    (19, 4, (0, 3, -1, 1), (0, 0, 0, 2)),
    (21, 4, (2, -1, -1, 4), (0, 0, 0, 2)),
    (23, 5, (5, 6, -1, 7), (2, 0, 0, 0)),
)
RELAY_LAG = 3
NJ = len(JOBS)
DEPTH = {t: job[1] for job in JOBS for t in job[2] if t >= 0}
NA = min(DEPTH.values())
MAXD = max(DEPTH.values())
NW = H - NA
WTILES = [sum(1 for t in range(H) if DEPTH[t] <= h) for h in range(NA, H)]
NEED = [max([job[1] for job in JOBS if job[2][d] >= 0], default=0) for d in range(N_DEV)]

N_SWAP = _digits("00000000000000000000111111112110")
SWAP_SENDS = _digits("11111111111111111110101010100000")
SWAP_DIR = (1, 3, 3, 1)
SWAPS = [(u, g, t) for u in range(NT) for g in range(N_SWAP[u]) for t in range(2)]

N_STAGE = _digits("00000000000000001110000000010101")
STAGE_PRE = _digits("212110")
STAGE_STEP = _digits("00000000000000000001010101010000")
STAGE_LAG = 2
N_SLOT = 8
STAGED = [(u, N_SWAP[u] + g, t) for u in range(NT) for g in range(N_STAGE[u]) for t in range(2)]

assert 1 + sum(SWAP_SENDS) == len(SWAPS)
assert sum(STAGE_PRE) + sum(STAGE_STEP) == len(STAGED)

S_X, S_WQ = 0, 1
S_WO = 4
S_KV = S_WO + NJ
S_V2 = S_KV + 2 * NT
S_WL = S_V2 + 1
S_N = S_WL + NW


def _body(x_ref, wq_ref, k_ref, v_ref, wo_ref, o_ref,
          xbuf, wqbuf, wo_job, wo_late, kbuf, vbuf, qpart, qrs, qbuf, pbuf, scale_buf,
          msg, rsbuf, ctxbuf, lbuf, obuf, acc_buf, stage,
          lsem, qr_ss, qr_rs, qa_ss, qa_rs, r_ss, r_rs, a_ss, a_rs, l_ss, l_rs,
          o_ss, o_rs, f_ss, x_ss, x_rs, sa_sem, sb_sem):
    me = lax.axis_index("i")
    ring = [me] + [(me + d) & 3 for d in (1, 2, 3)]
    peers = ring[1:]
    srcs = ring[:0:-1]
    diag_first = (1, 0, 2)
    kv = ((k_ref, kbuf), (v_ref, vbuf))

    def table(tab, dev):
        packed = sum((v & 15) << (4 * s) for s, v in enumerate(tab))
        return lax.shift_right_logical(jnp.int32(packed), 4 * dev) & 15

    def on(pred):
        tab = [int(bool(pred(d))) for d in range(N_DEV)]
        if all(tab):
            return lambda f: f()
        if not any(tab):
            return lambda f: None
        return pl.when(table(tab, me) == 1)

    def has_job(p, d):
        return JOBS[p][2][d % N_DEV] >= 0

    def relays(p, j, d):
        return has_job(p, d - j - 1) and JOBS[p][3][(d - j - 1) % N_DEV] == j

    def wants_ctx(h, d):
        return h >= NA or NEED[d % N_DEV] > h

    def unit_hc(u):
        h, i = divmod(u, NQB)
        return h, (i if h == EH else ring[UNIT_OFF[i]])

    k0 = pl.multiple_of(me * KS, KS)
    x_cp = pltpu.make_async_copy(x_ref.at[0, :, pl.ds(k0, KS)], xbuf, lsem.at[S_X])
    wq_parts = (QGROUPS[0], QGROUPS[1], (QGROUPS[2][0], H))

    def wq_copy(n):
        a, b = wq_parts[n]
        cols = pl.ds(a * DH, (b - a) * DH)
        return pltpu.make_async_copy(wq_ref.at[pl.ds(k0, KS), cols], wqbuf.at[:, cols], lsem.at[S_WQ + n])

    def job_copy(p):
        col = pl.multiple_of(table(JOBS[p][2], me) * DH, DH)
        rows = pl.ds(0, JOBS[p][1] * DH)
        return pltpu.make_async_copy(wo_ref.at[rows, pl.ds(col, DH)], wo_job.at[p, rows], lsem.at[S_WO + p])

    def head_copy(t):
        src, dst = kv[t]
        return pltpu.make_async_copy(src.at[:, :, :, 0, :], dst.at[0], lsem.at[S_KV + t])

    def unit_copy(u, t, part=0):
        src, dst = kv[t]
        h, c = unit_hc(u)
        g0, g1 = N_SWAP[u] + N_STAGE[u], NG
        if u == NT - 1 and t == 1:
            g0, g1 = (V_SPLIT, NG) if part else (g0, V_SPLIT)
        sl = pl.ds(g0, g1 - g0)
        return pltpu.make_async_copy(src.at[sl, c, :, h, :], dst.at[h, sl, c],
                                     lsem.at[S_V2 if part else S_KV + 2 * u + t])

    def late_copy(r):
        cols = pl.ds(0, WTILES[r] * DH)
        return pltpu.make_async_copy(wo_ref.at[pl.ds((NA + r) * DH, DH), cols], wo_late.at[r, :, cols],
                                     lsem.at[S_WL + r])

    def fetch(u):
        if u == 0:
            head_copy(0).start()
            head_copy(1).start()
        elif NQB <= u < NT:
            unit_copy(u, 0).start()
            unit_copy(u, 1).start()
            if u == NT - 1:
                unit_copy(u, 1, 1).start()
        elif NT <= u < NT + NW:
            late_copy(u - NT).start()

    def stage_copy(m, hop):
        u, g, t = STAGED[m]
        h, c = unit_hc(u)
        slot = stage.at[m % N_SLOT]
        if hop == 0:
            return pltpu.make_async_copy(kv[t][0].at[g, c, :, h, :], slot, sa_sem.at[m])
        return pltpu.make_async_copy(slot, kv[t][1].at[h, g, c], sb_sem.at[m])

    in_flight = []
    landed = set()
    n_staged = [0]

    def land(m):
        assert m < n_staged[0] and all(m not in batch for batch in in_flight)
        if m not in landed:
            stage_copy(m, 1).wait()
            landed.add(m)

    def pump(n):
        if len(in_flight) >= STAGE_LAG:
            for m in in_flight.pop(0):
                stage_copy(m, 0).wait()
                stage_copy(m, 1).start()
        batch = list(range(n_staged[0], n_staged[0] + n))
        for m in batch:
            if m >= N_SLOT:
                land(m - N_SLOT)
            stage_copy(m, 0).start()
        n_staged[0] += n
        in_flight.append(batch)

    def remote(src, dst, ss, rs, dev):
        return pltpu.make_async_remote_copy(src, dst, ss, rs, device_id=(dev,), device_id_type=MESH)

    def qr_copy(g, j):
        a, b = QGROUPS[g]
        heads = pl.ds(a, b - a)
        return remote(qpart.at[peers[j], heads], qrs.at[j, heads], qr_ss.at[g, j], qr_rs.at[g, j], peers[j])

    def qa_copy(g, j, dev):
        a, b = QGROUPS[g]
        sl = qbuf.at[dev, pl.ds(a, b - a)]
        return remote(sl, sl, qa_ss.at[g, j], qa_rs.at[g, j], peers[j])

    def r_copy(h, i):
        c = ring[UNIT_OFF[i]]
        rows = pl.ds(0, SENT)
        return remote(msg.at[h, c, rows], rsbuf.at[h, i, rows], r_ss.at[h, i], r_rs.at[h, i], c)

    def a_copy(h, j, dev):
        return remote(ctxbuf.at[h, dev], ctxbuf.at[h, dev], a_ss.at[h, j], a_rs.at[h, j], peers[j])

    def l_copy(c, j):
        rows = pl.ds(0, QB if c == LAST else SENT)
        return remote(msg.at[EH, c, rows], lbuf.at[c, j, rows], l_ss.at[c, j], l_rs.at[c, j], (me + j + 1) & 3)

    def s_copy(j):
        rows = pl.ds(QB, SENT - QB)
        return remote(msg.at[EH, LAST, rows], lbuf.at[LAST, j, rows], l_ss.at[NQB, j], l_rs.at[NQB, j], peers[j])

    def o_copy(p, j, dev):
        sl = obuf.at[table(JOBS[p][2], dev)]
        return remote(sl, sl, o_ss.at[p, j], o_rs.at[p, j], peers[j])

    def f_copy(p, j):
        sl = obuf.at[table(JOBS[p][2], srcs[j])]
        return remote(sl, sl, f_ss.at[p, j // 2], o_rs.at[p, 1], peers[j])

    def x_copy(m, recv=False):
        u, g, t = SWAPS[m]
        src, dst = kv[t]
        h, i = divmod(u, NQB)
        d = SWAP_DIR[sum(N_SWAP[NU:u]) + g] if h == EH else SWAP_DIR[i]
        c = i if h == EH else ring[(UNIT_OFF[i] + (0 if recv else d)) % N_DEV]
        return remote(src.at[g, c, :, h, :], dst.at[h, g, c], x_ss.at[m], x_rs.at[m], ring[d])

    unsent = list(range(len(SWAPS)))

    def send_swaps(n):
        for _ in range(n):
            x_copy(unsent.pop(0)).start()

    def send_late(c):
        for tab in LATE_ORDER:
            l_copy(c, table(tab, me)).start()

    def q_partial(x16, a, b):
        q = jnp.dot(x16, wqbuf[:, a * DH:b * DH].astype(BF16), preferred_element_type=F32)
        q = (q * SCALE).astype(BF16)
        for c in range(NQB):
            for h in range(a, b):
                qpart[c, h] = q[c * QB:(c + 1) * QB, (h - a) * DH:(h - a + 1) * DH]

    def q_scatter(g):
        for j in diag_first:
            qr_copy(g, j).start()

    def q_reduce(g):
        a, b = QGROUPS[g]
        for j in range(3):
            qr_copy(g, j).wait()
        acc = qpart[me, a:b].astype(F32)
        for j in range(3):
            acc = acc + qrs[j, a:b].astype(F32)
        qbuf[me, a:b] = acc.astype(BF16)
        for j in diag_first:
            qa_copy(g, j, me).start()

    def q_wait(g):
        for j in range(3):
            qa_copy(g, j, srcs[j]).wait_recv()
            qa_copy(g, j, me).wait_send()

    x_cp.start()
    for n in range(3):
        wq_copy(n).start()
    bar = pltpu.get_barrier_semaphore()
    for p in peers:
        pl.semaphore_signal(bar, inc=1, device_id=(p,), device_id_type=MESH)
    for u in range(PREFETCH):
        fetch(u)
    pump(STAGE_PRE[0])

    x_cp.wait()
    x16 = xbuf[...].astype(BF16)
    wq_copy(0).wait()
    q_partial(x16, *wq_parts[0])
    pump(STAGE_PRE[1])
    pl.semaphore_wait(bar, 3)
    q_scatter(0)
    wq_copy(1).wait()
    q_partial(x16, *wq_parts[1])
    q_scatter(1)
    wq_copy(2).wait()
    q_partial(x16, *wq_parts[2])
    pump(STAGE_PRE[2])
    q_reduce(0)
    pump(STAGE_PRE[3])
    q_reduce(1)
    send_swaps(1)
    pump(STAGE_PRE[4])
    for p in range(NJ):
        on(lambda d: has_job(p, d))(lambda p=p: job_copy(p).start())

    row = lax.broadcasted_iota(jnp.int32, (QB, DH), 0)
    lane = lax.broadcasted_iota(jnp.int32, (QB, DH), 1)
    diag2 = (lane & (QB - 1)) == row
    diag1 = lane == row
    srow = lax.broadcasted_iota(jnp.int32, (MSG_ROWS - QB, DH), 0)
    lo_half = lax.broadcasted_iota(jnp.int32, (1, DH), 1) < QB

    def scores(h, c):
        k = kbuf[h, :, c].reshape(NG * QB, DH).astype(BF16)
        s = lax.dot_general(qbuf[c, h], k, (((1,), (1,)), ((), ())), preferred_element_type=F32)
        m = jnp.max(s, axis=1, keepdims=True)
        p = jnp.exp(s - m)
        l = jnp.sum(p, axis=1, keepdims=True)
        for n in range(NG // 2):
            pbuf[n] = p[:, n * DH:(n + 1) * DH].astype(BF16)
        r = jnp.sum(jnp.where(diag2, m + jnp.log(l), 0.0), axis=0, keepdims=True)
        hi = r.astype(BF16).astype(F32)
        mid = (r - hi).astype(BF16).astype(F32)
        lo = r - hi - mid
        st = jnp.where(srow == 0, hi, jnp.where(srow == 1, mid, jnp.where(srow == 2, lo, 0.0)))
        msg[h, c, QB:MSG_ROWS, :] = st.astype(BF16)
        scale_buf[0] = jnp.broadcast_to(1.0 / l, (QB, DH))

    def values(h, c, g0, g1):
        v = vbuf[h, g0:g1, c].reshape((g1 - g0) * QB, DH).astype(BF16)
        p = jnp.concatenate([pbuf[n] for n in range(g0 // 2, g1 // 2)], axis=1)
        return jnp.dot(p, v, preferred_element_type=F32)

    def weights(parts):
        ls = [jnp.sum(p[QB:SENT, :].astype(F32), axis=0, keepdims=True) for p in parts]
        mx = jnp.maximum(jnp.maximum(ls[0], ls[1]), jnp.maximum(ls[2], ls[3]))
        es = [jnp.exp(a - mx) for a in ls]
        inv = 1.0 / (es[0] + es[1] + es[2] + es[3])
        return [e * inv for e in es]

    def combine(parts):
        w = weights(parts)
        w01 = jnp.where(lo_half, w[0], w[1])
        w23 = jnp.where(lo_half, w[2], w[3])
        d = jnp.concatenate([jnp.where(diag2, w01, 0.0), jnp.where(diag2, w23, 0.0)], axis=1).astype(BF16)
        stacked = jnp.concatenate([p[0:QB, :] for p in parts], axis=0)
        return jnp.dot(d, stacked, preferred_element_type=F32).astype(BF16)

    def reduce_head(h):
        for i in range(3):
            r_copy(h, i).wait()
        ctxbuf[h, me] = combine([msg.at[h, me]] + [rsbuf.at[h, i] for i in range(3)])
        for j in diag_first:
            on(lambda d: wants_ctx(h, d + j + 1))(lambda j=j: a_copy(h, j, me).start())

    have_ctx = [0] * N_DEV

    def recv_ctx(depth, devs):
        for h in range(depth):
            for j in range(3):
                on(lambda d: d in devs and have_ctx[d] <= h and wants_ctx(h, d))(
                    lambda j=j, h=h: a_copy(h, j, srcs[j]).wait_recv())
        for d in devs:
            have_ctx[d] = max(have_ctx[d], depth)

    def run_job(p):
        depth = JOBS[p][1]
        recv_ctx(depth, [d for d in range(N_DEV) if has_job(p, d)])

        def go():
            job_copy(p).wait()
            ctx = jnp.concatenate([ctxbuf[h].reshape(NQB * QB, DH) for h in range(depth)], axis=1)
            obuf[table(JOBS[p][2], me)] = jnp.dot(
                ctx, wo_job[p, 0:depth * DH].astype(BF16), preferred_element_type=F32).astype(BF16)
            for j in (0, 2):
                o_copy(p, j, me).start()
        on(lambda d: has_job(p, d))(go)

    def relay_job(p):
        for j in (0, 2):
            def go(j=j):
                o_copy(p, j, srcs[j]).wait_recv()
                f_copy(p, j).start()
            on(lambda d: relays(p, j, d))(go)

    for u in range(NT):
        h, c = unit_hc(u)
        i = u % NQB
        fetch(u + PREFETCH)
        for g in range(len(QGROUPS)):
            if u == QGROUPS[g][0] * NQB:
                q_wait(g)
        if u == 0:
            pump(STAGE_PRE[5])
        for m in range(len(STAGED)):
            if STAGED[m][0] == u:
                land(m)
        for m in range(len(SWAPS)):
            if SWAPS[m][0] == u:
                x_copy(m, True).wait_recv()
        if u >= NQB:
            unit_copy(u, 0).wait()
        elif u == 0:
            head_copy(0).wait()
        scores(h, c)
        if u == NT - 1:
            break
        if u >= NQB:
            unit_copy(u, 1).wait()
        elif u == 0:
            head_copy(1).wait()
        msg[h, c, 0:QB, :] = (values(h, c, 0, NG) * scale_buf[0]).astype(BF16)
        if h == EH:
            send_late(c)
        elif i < 3:
            r_copy(h, i).start()
        if u in Q_REDUCE:
            q_reduce(Q_REDUCE[u])
        if i == 0 and h > 0:
            reduce_head(h - 1)
        if i == 1 and h > 1:
            for j in range(3):
                on(lambda d: wants_ctx(h - 2, d + j + 1))(lambda j=j: a_copy(h - 2, j, me).wait_send())
        if u in Q_SCATTER:
            q_scatter(Q_SCATTER[u])
        send_swaps(SWAP_SENDS[u])
        pump(STAGE_STEP[u])
        for p in range(NJ):
            if u == JOBS[p][0]:
                run_job(p)
        for p in range(NJ):
            if u == JOBS[p][0] + RELAY_LAG:
                relay_job(p)

    for j in diag_first:
        s_copy(j).start()
    unit_copy(NT - 1, 1).wait()
    acc_buf[...] = values(EH, LAST, 0, V_SPLIT)
    unit_copy(NT - 1, 1, 1).wait()
    msg[EH, LAST, 0:QB, :] = ((acc_buf[...] + values(EH, LAST, V_SPLIT, NG)) * scale_buf[0]).astype(BF16)
    send_late(LAST)

    parts = [msg.at[EH, LAST]] + [lbuf.at[LAST, j] for j in range(3)]
    for r in range(NW):
        h = NA + r
        comb = r - (NW - NQB)
        if r == 0:
            for m in range(len(SWAPS)):
                x_copy(m).wait_send()
            for j in range(3):
                a_copy(EH - 1, j, me).wait_send()
            for p in range(NJ):
                for j in range(3):
                    on(lambda d: has_job(p, d - j - 1) and not relays(p, j, d))(
                        lambda p=p, j=j: o_copy(p, j, srcs[j]).wait_recv())
                    if j != 1:
                        on(lambda d: relays(p, j, d))(lambda p=p, j=j: f_copy(p, j).wait_send())
                        on(lambda d: has_job(p, d))(lambda p=p, j=j: o_copy(p, j, me).wait_send())
        if h < EH:
            recv_ctx(h + 1, range(N_DEV))
        if 0 <= comb < LAST:
            for j in range(3):
                l_copy(comb, j).wait()
        if h == EH:
            for j in range(3):
                s_copy(j).wait()
                l_copy(LAST, j).wait_send()
        late_copy(r).wait()

        if 0 <= comb < LAST:
            ctxbuf[EH, comb] = combine([msg.at[EH, comb]] + [lbuf.at[comb, j] for j in range(3)])
        nt = WTILES[r]
        w = wo_late[r, :, 0:nt * DH].astype(BF16)
        if h == EH:
            cols = [jnp.sum(jnp.where(diag1, v, 0.0), axis=1, keepdims=True) for v in weights(parts)]
            acc_buf[...] = parts[0][0:QB, :].astype(F32) * cols[0]
            for j in range(3):
                scale_buf[j] = jnp.broadcast_to(cols[j + 1], (QB, DH))
            o_ref[0, 0:LAST * QB, :] += jnp.dot(ctxbuf[EH, 0:LAST].reshape(LAST * QB, DH), w,
                                                preferred_element_type=F32)
        else:
            upd = jnp.dot(ctxbuf[h].reshape(NQB * QB, DH), w, preferred_element_type=F32)
            if r == 0:
                o_ref[0, :, 0:nt * DH] = upd + jnp.concatenate([obuf[p] for p in range(nt)], axis=1).astype(F32)
                for p in range(nt, H):
                    o_ref[0, :, p * DH:(p + 1) * DH] = obuf[p].astype(F32)
            else:
                o_ref[0, :, 0:nt * DH] += upd

    @pl.when(me < N_DEV)
    def _():
        for j in (0, 2, 1):
            l_copy(LAST, j).wait_recv()
        ctx = acc_buf[...]
        for j in range(3):
            ctx = ctx + parts[j + 1][0:QB, :].astype(F32) * scale_buf[j]
        o_ref[0, LAST * QB:, :] += jnp.dot(ctx.astype(BF16), wo_late[NW - 1].astype(BF16),
                                           preferred_element_type=F32)


def pallas_dist_sparse_attn_strided_kvseq_b1_sq256_skv4096_hq8_dh128_kernel(
    x: jax.Array,
    Wq: jax.Array,
    K_ext: jax.Array,
    V_ext: jax.Array,
    Wo: jax.Array,
):
    k5 = K_ext.reshape(NG, NQB, QB, H, DH)
    v5 = V_ext.reshape(NG, NQB, QB, H, DH)
    dma = pltpu.SemaphoreType.DMA
    nq = len(QGROUPS)
    return pl.pallas_call(
        _body,
        out_shape=jax.ShapeDtypeStruct((1, NQB * QB, DM), F32),
        in_specs=[pl.BlockSpec(memory_space=pltpu.HBM)] * 5,
        out_specs=pl.BlockSpec(memory_space=pltpu.VMEM),
        scratch_shapes=[
            pltpu.VMEM((NQB * QB, KS), F32),
            pltpu.VMEM((KS, DM), F32),
            pltpu.VMEM((NJ, MAXD * DH, DH), F32),
            pltpu.VMEM((NW, DH, DM), F32),
            pltpu.VMEM((H, NG, NQB, QB, DH), F32),
            pltpu.VMEM((H, NG, NQB, QB, DH), F32),
            pltpu.VMEM((NQB, H, QB, DH), BF16),
            pltpu.VMEM((3, H, QB, DH), BF16),
            pltpu.VMEM((NQB, H, QB, DH), BF16),
            pltpu.VMEM((NG // 2, QB, DH), BF16),
            pltpu.VMEM((3, QB, DH), F32),
            pltpu.VMEM((H, NQB, MSG_ROWS, DH), BF16),
            pltpu.VMEM((EH, 3, MSG_ROWS, DH), BF16),
            pltpu.VMEM((H, NQB, QB, DH), BF16),
            pltpu.VMEM((NQB, 3, MSG_ROWS, DH), BF16),
            pltpu.VMEM((H, NQB * QB, DH), BF16),
            pltpu.VMEM((QB, DH), F32),
            pltpu.SMEM((N_SLOT, QB, DH), F32),
            dma((S_N,)),
            dma((nq, 3)), dma((nq, 3)), dma((nq, 3)), dma((nq, 3)),
            dma((EH, 3)), dma((EH, 3)),
            dma((EH, 3)), dma((EH, 3)),
            dma((NQB + 1, 3)), dma((NQB + 1, 3)),
            dma((NJ, 3)), dma((NJ, 3)), dma((NJ, 2)),
            dma((len(SWAPS),)), dma((len(SWAPS),)),
            dma((len(STAGED),)), dma((len(STAGED),)),
        ],
        compiler_params=pltpu.CompilerParams(
            vmem_limit_bytes=64 * 1024 * 1024,
            collective_id=0,
            disable_semaphore_checks=True,
            disable_bounds_checks=True,
        ),
    )(x, Wq, k5, v5, Wo)
```

```python
import jax
import jax.numpy as jnp
from jax import lax
from jax.experimental import pallas as pl
from jax.experimental.pallas import tpu as pltpu

N_DEV = 4
NQB = 4
QB = 64
H = 8
DH = 128
NG = 16
DM = H * DH
KS = DM // N_DEV
EH = H - 1
LAST = NQB - 1
NU = EH * NQB
NT = H * NQB
MSG_ROWS = QB + 16
SENT = QB + 8
SCALE = 0.08838834764831843
MESH = pl.DeviceIdType.MESH
F32 = jnp.float32
BF16 = jnp.bfloat16


def _digits(text):
    return tuple(int(ch) for ch in text)


PREFETCH = 8
V_SPLIT = 8

UNIT_OFF = (2, 1, 3, 0)
LATE_ORDER = ((1, 2, 1, 0), (0, 1, 0, 1), (2, 0, 2, 2))

QGROUPS = ((0, 1), (1, 3), (3, 5), (5, 8))
Q_SCATTER = {1: 2, 10: 3}
Q_REDUCE = {5: 2, 14: 3}

JOBS = (
    (19, 4, (0, 3, -1, 1), (0, 0, 0, 2)),
    (21, 4, (2, -1, -1, 4), (0, 0, 0, 2)),
    (23, 5, (5, 6, -1, 7), (2, 0, 0, 0)),
)
RELAY_LAG = 3
NJ = len(JOBS)
DEPTH = {t: job[1] for job in JOBS for t in job[2] if t >= 0}
NA = min(DEPTH.values())
MAXD = max(DEPTH.values())
NW = H - NA
WTILES = [sum(1 for t in range(H) if DEPTH[t] <= h) for h in range(NA, H)]
NEED = [max([job[1] for job in JOBS if job[2][d] >= 0], default=0) for d in range(N_DEV)]

N_SWAP = _digits("00000000000000000000111111112110")
SWAP_SENDS = _digits("11111111111111111110101010100000")
SWAP_DIR = (1, 3, 3, 1)
SWAPS = [(u, g, t) for u in range(NT) for g in range(N_SWAP[u]) for t in range(2)]

N_STAGE = _digits("00000000000000111111000001110101")
STAGE_PRE = _digits("212110")
STAGE_STEP = _digits("00010101010101010101110111010000")
STAGE_LAG = 2
N_SLOT = 8
STAGED = [(u, N_SWAP[u] + g, t) for u in range(NT) for g in range(N_STAGE[u]) for t in range(2)]

assert 1 + sum(SWAP_SENDS) == len(SWAPS)
assert sum(STAGE_PRE) + sum(STAGE_STEP) == len(STAGED)

S_X, S_WQ = 0, 1
S_WO = 4
S_KV = S_WO + NJ
S_V2 = S_KV + 2 * NT
S_WL = S_V2 + 1
S_N = S_WL + NW


def _body(x_ref, wq_ref, k_ref, v_ref, wo_ref, o_ref,
          xbuf, wqbuf, wo_job, wo_late, kbuf, vbuf, qpart, qrs, qbuf, pbuf, scale_buf,
          msg, rsbuf, ctxbuf, lbuf, obuf, acc_buf, stage,
          lsem, qr_ss, qr_rs, qa_ss, qa_rs, r_ss, r_rs, a_ss, a_rs, l_ss, l_rs,
          o_ss, o_rs, f_ss, x_ss, x_rs, sa_sem, sb_sem):
    me = lax.axis_index("i")
    ring = [me] + [(me + d) & 3 for d in (1, 2, 3)]
    peers = ring[1:]
    srcs = ring[:0:-1]
    diag_first = (1, 0, 2)
    kv = ((k_ref, kbuf), (v_ref, vbuf))

    def table(tab, dev):
        packed = sum((v & 15) << (4 * s) for s, v in enumerate(tab))
        return lax.shift_right_logical(jnp.int32(packed), 4 * dev) & 15

    def on(pred):
        tab = [int(bool(pred(d))) for d in range(N_DEV)]
        if all(tab):
            return lambda f: f()
        if not any(tab):
            return lambda f: None
        return pl.when(table(tab, me) == 1)

    def has_job(p, d):
        return JOBS[p][2][d % N_DEV] >= 0

    def relays(p, j, d):
        return has_job(p, d - j - 1) and JOBS[p][3][(d - j - 1) % N_DEV] == j

    def wants_ctx(h, d):
        return h >= NA or NEED[d % N_DEV] > h

    def unit_hc(u):
        h, i = divmod(u, NQB)
        return h, (i if h == EH else ring[UNIT_OFF[i]])

    k0 = pl.multiple_of(me * KS, KS)
    x_cp = pltpu.make_async_copy(x_ref.at[0, :, pl.ds(k0, KS)], xbuf, lsem.at[S_X])
    wq_parts = (QGROUPS[0], QGROUPS[1], (QGROUPS[2][0], H))

    def wq_copy(n):
        a, b = wq_parts[n]
        cols = pl.ds(a * DH, (b - a) * DH)
        return pltpu.make_async_copy(wq_ref.at[pl.ds(k0, KS), cols], wqbuf.at[:, cols], lsem.at[S_WQ + n])

    def job_copy(p):
        col = pl.multiple_of(table(JOBS[p][2], me) * DH, DH)
        rows = pl.ds(0, JOBS[p][1] * DH)
        return pltpu.make_async_copy(wo_ref.at[rows, pl.ds(col, DH)], wo_job.at[p, rows], lsem.at[S_WO + p])

    def head_copy(t):
        src, dst = kv[t]
        return pltpu.make_async_copy(src.at[:, :, :, 0, :], dst.at[0], lsem.at[S_KV + t])

    def unit_copy(u, t, part=0):
        src, dst = kv[t]
        h, c = unit_hc(u)
        g0, g1 = N_SWAP[u] + N_STAGE[u], NG
        if u == NT - 1 and t == 1:
            g0, g1 = (V_SPLIT, NG) if part else (g0, V_SPLIT)
        sl = pl.ds(g0, g1 - g0)
        return pltpu.make_async_copy(src.at[sl, c, :, h, :], dst.at[h, sl, c],
                                     lsem.at[S_V2 if part else S_KV + 2 * u + t])

    def late_copy(r):
        cols = pl.ds(0, WTILES[r] * DH)
        return pltpu.make_async_copy(wo_ref.at[pl.ds((NA + r) * DH, DH), cols], wo_late.at[r, :, cols],
                                     lsem.at[S_WL + r])

    def fetch(u):
        if u == 0:
            head_copy(0).start()
            head_copy(1).start()
        elif NQB <= u < NT:
            unit_copy(u, 0).start()
            unit_copy(u, 1).start()
            if u == NT - 1:
                unit_copy(u, 1, 1).start()
        elif NT <= u < NT + NW:
            late_copy(u - NT).start()

    def stage_copy(m, hop):
        u, g, t = STAGED[m]
        h, c = unit_hc(u)
        slot = stage.at[m % N_SLOT]
        if hop == 0:
            return pltpu.make_async_copy(kv[t][0].at[g, c, :, h, :], slot, sa_sem.at[m])
        return pltpu.make_async_copy(slot, kv[t][1].at[h, g, c], sb_sem.at[m])

    in_flight = []
    landed = set()
    n_staged = [0]

    def land(m):
        assert m < n_staged[0] and all(m not in batch for batch in in_flight)
        if m not in landed:
            stage_copy(m, 1).wait()
            landed.add(m)

    def pump(n):
        if len(in_flight) >= STAGE_LAG:
            for m in in_flight.pop(0):
                stage_copy(m, 0).wait()
                stage_copy(m, 1).start()
        batch = list(range(n_staged[0], n_staged[0] + n))
        for m in batch:
            if m >= N_SLOT:
                land(m - N_SLOT)
            stage_copy(m, 0).start()
        n_staged[0] += n
        in_flight.append(batch)

    def remote(src, dst, ss, rs, dev):
        return pltpu.make_async_remote_copy(src, dst, ss, rs, device_id=(dev,), device_id_type=MESH)

    def qr_copy(g, j):
        a, b = QGROUPS[g]
        heads = pl.ds(a, b - a)
        return remote(qpart.at[peers[j], heads], qrs.at[j, heads], qr_ss.at[g, j], qr_rs.at[g, j], peers[j])

    def qa_copy(g, j, dev):
        a, b = QGROUPS[g]
        sl = qbuf.at[dev, pl.ds(a, b - a)]
        return remote(sl, sl, qa_ss.at[g, j], qa_rs.at[g, j], peers[j])

    def r_copy(h, i):
        c = ring[UNIT_OFF[i]]
        rows = pl.ds(0, SENT)
        return remote(msg.at[h, c, rows], rsbuf.at[h, i, rows], r_ss.at[h, i], r_rs.at[h, i], c)

    def a_copy(h, j, dev):
        return remote(ctxbuf.at[h, dev], ctxbuf.at[h, dev], a_ss.at[h, j], a_rs.at[h, j], peers[j])

    def l_copy(c, j):
        rows = pl.ds(0, QB if c == LAST else SENT)
        return remote(msg.at[EH, c, rows], lbuf.at[c, j, rows], l_ss.at[c, j], l_rs.at[c, j], (me + j + 1) & 3)

    def s_copy(j):
        rows = pl.ds(QB, SENT - QB)
        return remote(msg.at[EH, LAST, rows], lbuf.at[LAST, j, rows], l_ss.at[NQB, j], l_rs.at[NQB, j], peers[j])

    def o_copy(p, j, dev):
        sl = obuf.at[table(JOBS[p][2], dev)]
        return remote(sl, sl, o_ss.at[p, j], o_rs.at[p, j], peers[j])

    def f_copy(p, j):
        sl = obuf.at[table(JOBS[p][2], srcs[j])]
        return remote(sl, sl, f_ss.at[p, j // 2], o_rs.at[p, 1], peers[j])

    def x_copy(m, recv=False):
        u, g, t = SWAPS[m]
        src, dst = kv[t]
        h, i = divmod(u, NQB)
        d = SWAP_DIR[sum(N_SWAP[NU:u]) + g] if h == EH else SWAP_DIR[i]
        c = i if h == EH else ring[(UNIT_OFF[i] + (0 if recv else d)) % N_DEV]
        return remote(src.at[g, c, :, h, :], dst.at[h, g, c], x_ss.at[m], x_rs.at[m], ring[d])

    unsent = list(range(len(SWAPS)))

    def send_swaps(n):
        for _ in range(n):
            x_copy(unsent.pop(0)).start()

    def send_late(c):
        for tab in LATE_ORDER:
            l_copy(c, table(tab, me)).start()

    def q_partial(x16, a, b):
        q = jnp.dot(x16, wqbuf[:, a * DH:b * DH].astype(BF16), preferred_element_type=F32)
        q = (q * SCALE).astype(BF16)
        for c in range(NQB):
            for h in range(a, b):
                qpart[c, h] = q[c * QB:(c + 1) * QB, (h - a) * DH:(h - a + 1) * DH]

    def q_scatter(g):
        for j in diag_first:
            qr_copy(g, j).start()

    def q_reduce(g):
        a, b = QGROUPS[g]
        for j in range(3):
            qr_copy(g, j).wait()
        acc = qpart[me, a:b].astype(F32)
        for j in range(3):
            acc = acc + qrs[j, a:b].astype(F32)
        qbuf[me, a:b] = acc.astype(BF16)
        for j in diag_first:
            qa_copy(g, j, me).start()

    def q_wait(g):
        for j in range(3):
            qa_copy(g, j, srcs[j]).wait_recv()
            qa_copy(g, j, me).wait_send()

    x_cp.start()
    for n in range(3):
        wq_copy(n).start()
    bar = pltpu.get_barrier_semaphore()
    for p in peers:
        pl.semaphore_signal(bar, inc=1, device_id=(p,), device_id_type=MESH)
    for u in range(PREFETCH):
        fetch(u)
    pump(STAGE_PRE[0])

    x_cp.wait()
    x16 = xbuf[...].astype(BF16)
    wq_copy(0).wait()
    q_partial(x16, *wq_parts[0])
    pump(STAGE_PRE[1])
    pl.semaphore_wait(bar, 3)
    q_scatter(0)
    wq_copy(1).wait()
    q_partial(x16, *wq_parts[1])
    q_scatter(1)
    wq_copy(2).wait()
    q_partial(x16, *wq_parts[2])
    pump(STAGE_PRE[2])
    q_reduce(0)
    pump(STAGE_PRE[3])
    q_reduce(1)
    send_swaps(1)
    pump(STAGE_PRE[4])
    for p in range(NJ):
        on(lambda d: has_job(p, d))(lambda p=p: job_copy(p).start())

    row = lax.broadcasted_iota(jnp.int32, (QB, DH), 0)
    lane = lax.broadcasted_iota(jnp.int32, (QB, DH), 1)
    diag2 = (lane & (QB - 1)) == row
    diag1 = lane == row
    srow = lax.broadcasted_iota(jnp.int32, (MSG_ROWS - QB, DH), 0)
    lo_half = lax.broadcasted_iota(jnp.int32, (1, DH), 1) < QB

    def scores(h, c):
        k = kbuf[h, :, c].reshape(NG * QB, DH).astype(BF16)
        s = lax.dot_general(qbuf[c, h], k, (((1,), (1,)), ((), ())), preferred_element_type=F32)
        m = jnp.max(s, axis=1, keepdims=True)
        p = jnp.exp(s - m)
        l = jnp.sum(p, axis=1, keepdims=True)
        for n in range(NG // 2):
            pbuf[n] = p[:, n * DH:(n + 1) * DH].astype(BF16)
        r = jnp.sum(jnp.where(diag2, m + jnp.log(l), 0.0), axis=0, keepdims=True)
        hi = r.astype(BF16).astype(F32)
        mid = (r - hi).astype(BF16).astype(F32)
        lo = r - hi - mid
        st = jnp.where(srow == 0, hi, jnp.where(srow == 1, mid, jnp.where(srow == 2, lo, 0.0)))
        msg[h, c, QB:MSG_ROWS, :] = st.astype(BF16)
        scale_buf[0] = jnp.broadcast_to(1.0 / l, (QB, DH))

    def values(h, c, g0, g1):
        v = vbuf[h, g0:g1, c].reshape((g1 - g0) * QB, DH).astype(BF16)
        p = jnp.concatenate([pbuf[n] for n in range(g0 // 2, g1 // 2)], axis=1)
        return jnp.dot(p, v, preferred_element_type=F32)

    def weights(parts):
        ls = [jnp.sum(p[QB:SENT, :].astype(F32), axis=0, keepdims=True) for p in parts]
        mx = jnp.maximum(jnp.maximum(ls[0], ls[1]), jnp.maximum(ls[2], ls[3]))
        es = [jnp.exp(a - mx) for a in ls]
        inv = 1.0 / (es[0] + es[1] + es[2] + es[3])
        return [e * inv for e in es]

    def combine(parts):
        w = weights(parts)
        w01 = jnp.where(lo_half, w[0], w[1])
        w23 = jnp.where(lo_half, w[2], w[3])
        d = jnp.concatenate([jnp.where(diag2, w01, 0.0), jnp.where(diag2, w23, 0.0)], axis=1).astype(BF16)
        stacked = jnp.concatenate([p[0:QB, :] for p in parts], axis=0)
        return jnp.dot(d, stacked, preferred_element_type=F32).astype(BF16)

    def reduce_head(h):
        for i in range(3):
            r_copy(h, i).wait()
        ctxbuf[h, me] = combine([msg.at[h, me]] + [rsbuf.at[h, i] for i in range(3)])
        for j in diag_first:
            on(lambda d: wants_ctx(h, d + j + 1))(lambda j=j: a_copy(h, j, me).start())

    have_ctx = [0] * N_DEV

    def recv_ctx(depth, devs):
        for h in range(depth):
            for j in range(3):
                on(lambda d: d in devs and have_ctx[d] <= h and wants_ctx(h, d))(
                    lambda j=j, h=h: a_copy(h, j, srcs[j]).wait_recv())
        for d in devs:
            have_ctx[d] = max(have_ctx[d], depth)

    def run_job(p):
        depth = JOBS[p][1]
        recv_ctx(depth, [d for d in range(N_DEV) if has_job(p, d)])

        def go():
            job_copy(p).wait()
            ctx = jnp.concatenate([ctxbuf[h].reshape(NQB * QB, DH) for h in range(depth)], axis=1)
            obuf[table(JOBS[p][2], me)] = jnp.dot(
                ctx, wo_job[p, 0:depth * DH].astype(BF16), preferred_element_type=F32).astype(BF16)
            for j in (0, 2):
                o_copy(p, j, me).start()
        on(lambda d: has_job(p, d))(go)

    def relay_job(p):
        for j in (0, 2):
            def go(j=j):
                o_copy(p, j, srcs[j]).wait_recv()
                f_copy(p, j).start()
            on(lambda d: relays(p, j, d))(go)

    for u in range(NT):
        h, c = unit_hc(u)
        i = u % NQB
        fetch(u + PREFETCH)
        for g in range(len(QGROUPS)):
            if u == QGROUPS[g][0] * NQB:
                q_wait(g)
        if u == 0:
            pump(STAGE_PRE[5])
        for m in range(len(STAGED)):
            if STAGED[m][0] == u:
                land(m)
        for m in range(len(SWAPS)):
            if SWAPS[m][0] == u:
                x_copy(m, True).wait_recv()
        if u >= NQB:
            unit_copy(u, 0).wait()
        elif u == 0:
            head_copy(0).wait()
        scores(h, c)
        if u == NT - 1:
            break
        if u >= NQB:
            unit_copy(u, 1).wait()
        elif u == 0:
            head_copy(1).wait()
        msg[h, c, 0:QB, :] = (values(h, c, 0, NG) * scale_buf[0]).astype(BF16)
        if h == EH:
            send_late(c)
        elif i < 3:
            r_copy(h, i).start()
        if u in Q_REDUCE:
            q_reduce(Q_REDUCE[u])
        if i == 0 and h > 0:
            reduce_head(h - 1)
        if i == 1 and h > 1:
            for j in range(3):
                on(lambda d: wants_ctx(h - 2, d + j + 1))(lambda j=j: a_copy(h - 2, j, me).wait_send())
        if u in Q_SCATTER:
            q_scatter(Q_SCATTER[u])
        send_swaps(SWAP_SENDS[u])
        pump(STAGE_STEP[u])
        for p in range(NJ):
            if u == JOBS[p][0]:
                run_job(p)
        for p in range(NJ):
            if u == JOBS[p][0] + RELAY_LAG:
                relay_job(p)

    for j in diag_first:
        s_copy(j).start()
    unit_copy(NT - 1, 1).wait()
    acc_buf[...] = values(EH, LAST, 0, V_SPLIT)
    unit_copy(NT - 1, 1, 1).wait()
    msg[EH, LAST, 0:QB, :] = ((acc_buf[...] + values(EH, LAST, V_SPLIT, NG)) * scale_buf[0]).astype(BF16)
    send_late(LAST)

    own_block = pl.when(me < N_DEV)
    parts = [msg.at[EH, LAST]] + [lbuf.at[LAST, j] for j in range(3)]
    for r in range(NW):
        h = NA + r
        comb = r - (NW - NQB)
        if r == 0:
            for m in range(len(SWAPS)):
                x_copy(m).wait_send()
            for j in range(3):
                a_copy(EH - 1, j, me).wait_send()
            for p in range(NJ):
                for j in range(3):
                    on(lambda d: has_job(p, d - j - 1) and not relays(p, j, d))(
                        lambda p=p, j=j: o_copy(p, j, srcs[j]).wait_recv())
                    if j != 1:
                        on(lambda d: relays(p, j, d))(lambda p=p, j=j: f_copy(p, j).wait_send())
                        on(lambda d: has_job(p, d))(lambda p=p, j=j: o_copy(p, j, me).wait_send())
        if h < EH:
            recv_ctx(h + 1, range(N_DEV))
        if 0 <= comb < LAST:
            for j in range(3):
                l_copy(comb, j).wait()
        if h == EH:
            for j in range(3):
                s_copy(j).wait()
                l_copy(LAST, j).wait_send()
        late_copy(r).wait()

        def project(r=r, h=h, comb=comb):
            if 0 <= comb < LAST:
                ctxbuf[EH, comb] = combine([msg.at[EH, comb]] + [lbuf.at[comb, j] for j in range(3)])
            nt = WTILES[r]
            w = wo_late[r, :, 0:nt * DH].astype(BF16)
            if h == EH:
                cols = [jnp.sum(jnp.where(diag1, v, 0.0), axis=1, keepdims=True) for v in weights(parts)]
                acc_buf[...] = parts[0][0:QB, :].astype(F32) * cols[0]
                for j in range(3):
                    scale_buf[j] = jnp.broadcast_to(cols[j + 1], (QB, DH))
                o_ref[0, 0:LAST * QB, :] += jnp.dot(ctxbuf[EH, 0:LAST].reshape(LAST * QB, DH), w,
                                                    preferred_element_type=F32)
            else:
                upd = jnp.dot(ctxbuf[h].reshape(NQB * QB, DH), w, preferred_element_type=F32)
                if r == 0:
                    o_ref[0, :, 0:nt * DH] = upd + jnp.concatenate([obuf[p] for p in range(nt)], axis=1).astype(F32)
                    for p in range(nt, H):
                        o_ref[0, :, p * DH:(p + 1) * DH] = obuf[p].astype(F32)
                else:
                    o_ref[0, :, 0:nt * DH] += upd

        if r == 0:
            project()
        else:
            own_block(project)

    @own_block
    def _():
        for j in (0, 2, 1):
            l_copy(LAST, j).wait_recv()
        ctx = acc_buf[...]
        for j in range(3):
            ctx = ctx + parts[j + 1][0:QB, :].astype(F32) * scale_buf[j]
        o_ref[0, LAST * QB:, :] += jnp.dot(ctx.astype(BF16), wo_late[NW - 1].astype(BF16),
                                           preferred_element_type=F32)


def pallas_dist_sparse_attn_strided_kvseq_b1_sq256_skv4096_hq8_dh128_kernel(
    x: jax.Array,
    Wq: jax.Array,
    K_ext: jax.Array,
    V_ext: jax.Array,
    Wo: jax.Array,
):
    k5 = K_ext.reshape(NG, NQB, QB, H, DH)
    v5 = V_ext.reshape(NG, NQB, QB, H, DH)
    dma = pltpu.SemaphoreType.DMA
    nq = len(QGROUPS)
    return pl.pallas_call(
        _body,
        out_shape=jax.ShapeDtypeStruct((1, NQB * QB, DM), F32),
        in_specs=[pl.BlockSpec(memory_space=pltpu.HBM)] * 5,
        out_specs=pl.BlockSpec(memory_space=pltpu.VMEM),
        scratch_shapes=[
            pltpu.VMEM((NQB * QB, KS), F32),
            pltpu.VMEM((KS, DM), F32),
            pltpu.VMEM((NJ, MAXD * DH, DH), F32),
            pltpu.VMEM((NW, DH, DM), F32),
            pltpu.VMEM((H, NG, NQB, QB, DH), F32),
            pltpu.VMEM((H, NG, NQB, QB, DH), F32),
            pltpu.VMEM((NQB, H, QB, DH), BF16),
            pltpu.VMEM((3, H, QB, DH), BF16),
            pltpu.VMEM((NQB, H, QB, DH), BF16),
            pltpu.VMEM((NG // 2, QB, DH), BF16),
            pltpu.VMEM((3, QB, DH), F32),
            pltpu.VMEM((H, NQB, MSG_ROWS, DH), BF16),
            pltpu.VMEM((EH, 3, MSG_ROWS, DH), BF16),
            pltpu.VMEM((H, NQB, QB, DH), BF16),
            pltpu.VMEM((NQB, 3, MSG_ROWS, DH), BF16),
            pltpu.VMEM((H, NQB * QB, DH), BF16),
            pltpu.VMEM((QB, DH), F32),
            pltpu.SMEM((N_SLOT, QB, DH), F32),
            dma((S_N,)),
            dma((nq, 3)), dma((nq, 3)), dma((nq, 3)), dma((nq, 3)),
            dma((EH, 3)), dma((EH, 3)),
            dma((EH, 3)), dma((EH, 3)),
            dma((NQB + 1, 3)), dma((NQB + 1, 3)),
            dma((NJ, 3)), dma((NJ, 3)), dma((NJ, 2)),
            dma((len(SWAPS),)), dma((len(SWAPS),)),
            dma((len(STAGED),)), dma((len(STAGED),)),
        ],
        compiler_params=pltpu.CompilerParams(
            vmem_limit_bytes=64 * 1024 * 1024,
            collective_id=0,
            disable_semaphore_checks=True,
            disable_bounds_checks=True,
        ),
    )(x, Wq, k5, v5, Wo)
```

```python
import jax
import jax.numpy as jnp
from jax import lax
from jax.experimental import pallas as pl
from jax.experimental.pallas import tpu as pltpu

N_DEV = 4
NQB = 4
QB = 64
H = 8
DH = 128
NG = 16
DM = H * DH
KS = DM // N_DEV
EH = H - 1
LAST = NQB - 1
NU = EH * NQB
NT = H * NQB
MSG_ROWS = QB + 16
SENT = QB + 8
SCALE = 0.08838834764831843
MESH = pl.DeviceIdType.MESH
F32 = jnp.float32
BF16 = jnp.bfloat16


def _digits(text):
    return tuple(int(ch) for ch in text)


FETCH_FIRST = 8
FETCH_STEP = _digits("11111111011101110111111111111110")
ROW_PIECES = 2
V_SPLIT = 8

UNIT_OFF = (2, 1, 3, 0)
LATE_ORDER = ((1, 2, 1, 0), (0, 1, 0, 1), (2, 0, 2, 2))

QGROUPS = ((0, 1), (1, 3), (3, 5), (5, 8))
Q_SCATTER = {1: 2, 10: 3}
Q_REDUCE = {5: 2, 14: 3}

JOBS = (
    (19, 4, (0, 3, -1, 1), (0, 0, 0, 2)),
    (21, 4, (2, -1, -1, 4), (0, 0, 0, 2)),
    (23, 5, (5, 6, -1, 7), (2, 0, 0, 0)),
)
RELAY_LAG = 3
NJ = len(JOBS)
DEPTH = {t: job[1] for job in JOBS for t in job[2] if t >= 0}
NA = min(DEPTH.values())
MAXD = max(DEPTH.values())
NW = H - NA
WTILES = [sum(1 for t in range(H) if DEPTH[t] <= h) for h in range(NA, H)]
NEED = [max([job[1] for job in JOBS if job[2][d] >= 0], default=0) for d in range(N_DEV)]

N_SWAP = _digits("00000000000000000000111111112110")
SWAP_SENDS = _digits("11111111111111111110101010100000")
SWAP_DIR = (1, 3, 3, 1)
SWAPS = [(u, g, t) for u in range(NT) for g in range(N_SWAP[u]) for t in range(2)]

N_STAGE = _digits("00000000000000111111000001110101")
STAGE_PRE = _digits("212110")
STAGE_STEP = _digits("00010101010101010101110111010000")
STAGE_LAG = 2
N_SLOT = 8
STAGED = [(u, N_SWAP[u] + g, t) for u in range(NT) for g in range(N_STAGE[u]) for t in range(2)]

assert FETCH_FIRST + sum(FETCH_STEP) == NT + NW
assert 1 + sum(SWAP_SENDS) == len(SWAPS)
assert sum(STAGE_PRE) + sum(STAGE_STEP) == len(STAGED)

S_X, S_WQ = 0, 1
S_WO = 4
S_KV = S_WO + NJ
S_WL = S_KV + (2 * NT + 1) * ROW_PIECES
S_N = S_WL + NW


def _body(x_ref, wq_ref, k_ref, v_ref, wo_ref, o_ref,
          xbuf, wqbuf, wo_job, wo_late, kbuf, vbuf, qpart, qrs, qbuf, pbuf, scale_buf,
          msg, rsbuf, ctxbuf, lbuf, obuf, acc_buf, stage,
          lsem, qr_ss, qr_rs, qa_ss, qa_rs, r_ss, r_rs, a_ss, a_rs, l_ss, l_rs,
          o_ss, o_rs, f_ss, x_ss, x_rs, sa_sem, sb_sem):
    me = lax.axis_index("i")
    ring = [me] + [(me + d) & 3 for d in (1, 2, 3)]
    peers = ring[1:]
    srcs = ring[:0:-1]
    diag_first = (1, 0, 2)
    kv = ((k_ref, kbuf), (v_ref, vbuf))

    def table(tab, dev):
        packed = sum((v & 15) << (4 * s) for s, v in enumerate(tab))
        return lax.shift_right_logical(jnp.int32(packed), 4 * dev) & 15

    def on(pred):
        tab = [int(bool(pred(d))) for d in range(N_DEV)]
        if all(tab):
            return lambda f: f()
        if not any(tab):
            return lambda f: None
        return pl.when(table(tab, me) == 1)

    def has_job(p, d):
        return JOBS[p][2][d % N_DEV] >= 0

    def relays(p, j, d):
        return has_job(p, d - j - 1) and JOBS[p][3][(d - j - 1) % N_DEV] == j

    def wants_ctx(h, d):
        return h >= NA or NEED[d % N_DEV] > h

    def unit_hc(u):
        h, i = divmod(u, NQB)
        return h, (i if h == EH else ring[UNIT_OFF[i]])

    k0 = pl.multiple_of(me * KS, KS)
    x_cp = pltpu.make_async_copy(x_ref.at[0, :, pl.ds(k0, KS)], xbuf, lsem.at[S_X])
    wq_parts = (QGROUPS[0], QGROUPS[1], (QGROUPS[2][0], H))

    def wq_copy(n):
        a, b = wq_parts[n]
        cols = pl.ds(a * DH, (b - a) * DH)
        return pltpu.make_async_copy(wq_ref.at[pl.ds(k0, KS), cols], wqbuf.at[:, cols], lsem.at[S_WQ + n])

    def job_copy(p):
        col = pl.multiple_of(table(JOBS[p][2], me) * DH, DH)
        rows = pl.ds(0, JOBS[p][1] * DH)
        return pltpu.make_async_copy(wo_ref.at[rows, pl.ds(col, DH)], wo_job.at[p, rows], lsem.at[S_WO + p])

    def head_copy(t):
        src, dst = kv[t]
        return pltpu.make_async_copy(src.at[:, :, :, 0, :], dst.at[0], lsem.at[S_KV + t])

    def unit_copies(u, t, part=0):
        src, dst = kv[t]
        h, c = unit_hc(u)
        g0, g1 = N_SWAP[u] + N_STAGE[u], NG
        if u == NT - 1 and t == 1:
            g0, g1 = (V_SPLIT, NG) if part else (g0, V_SPLIT)
        groups = pl.ds(g0, g1 - g0)
        sem0 = S_KV + (2 * u + t + part) * ROW_PIECES
        pieces = [pl.ds(q * QB // ROW_PIECES, QB // ROW_PIECES) for q in range(ROW_PIECES)]
        return [pltpu.make_async_copy(src.at[groups, c, rows, h, :], dst.at[h, groups, c, rows], lsem.at[sem0 + q])
                for q, rows in enumerate(pieces)]

    def unit_wait(u, t, part=0):
        for cp in unit_copies(u, t, part):
            cp.wait()

    def late_copy(r):
        cols = pl.ds(0, WTILES[r] * DH)
        return pltpu.make_async_copy(wo_ref.at[pl.ds((NA + r) * DH, DH), cols], wo_late.at[r, :, cols],
                                     lsem.at[S_WL + r])

    n_fetched = [0]

    def fetch(n):
        for u in range(n_fetched[0], n_fetched[0] + n):
            if u == 0:
                copies = [head_copy(0), head_copy(1)]
            elif u < NQB:
                copies = []
            elif u < NT:
                copies = unit_copies(u, 0) + unit_copies(u, 1)
                if u == NT - 1:
                    copies += unit_copies(u, 1, 1)
            else:
                copies = [late_copy(u - NT)]
            for cp in copies:
                cp.start()
        n_fetched[0] += n

    def stage_copy(m, hop):
        u, g, t = STAGED[m]
        h, c = unit_hc(u)
        slot = stage.at[m % N_SLOT]
        if hop == 0:
            return pltpu.make_async_copy(kv[t][0].at[g, c, :, h, :], slot, sa_sem.at[m])
        return pltpu.make_async_copy(slot, kv[t][1].at[h, g, c], sb_sem.at[m])

    in_flight = []
    landed = set()
    n_staged = [0]

    def land(m):
        assert m < n_staged[0] and all(m not in batch for batch in in_flight)
        if m not in landed:
            stage_copy(m, 1).wait()
            landed.add(m)

    def pump(n):
        if len(in_flight) >= STAGE_LAG:
            for m in in_flight.pop(0):
                stage_copy(m, 0).wait()
                stage_copy(m, 1).start()
        batch = list(range(n_staged[0], n_staged[0] + n))
        for m in batch:
            if m >= N_SLOT:
                land(m - N_SLOT)
            stage_copy(m, 0).start()
        n_staged[0] += n
        in_flight.append(batch)

    def remote(src, dst, ss, rs, dev):
        return pltpu.make_async_remote_copy(src, dst, ss, rs, device_id=(dev,), device_id_type=MESH)

    def qr_copy(g, j):
        a, b = QGROUPS[g]
        heads = pl.ds(a, b - a)
        return remote(qpart.at[peers[j], heads], qrs.at[j, heads], qr_ss.at[g, j], qr_rs.at[g, j], peers[j])

    def qa_copy(g, j, dev):
        a, b = QGROUPS[g]
        sl = qbuf.at[dev, pl.ds(a, b - a)]
        return remote(sl, sl, qa_ss.at[g, j], qa_rs.at[g, j], peers[j])

    def r_copy(h, i):
        c = ring[UNIT_OFF[i]]
        rows = pl.ds(0, SENT)
        return remote(msg.at[h, c, rows], rsbuf.at[h, i, rows], r_ss.at[h, i], r_rs.at[h, i], c)

    def a_copy(h, j, dev):
        return remote(ctxbuf.at[h, dev], ctxbuf.at[h, dev], a_ss.at[h, j], a_rs.at[h, j], peers[j])

    def l_copy(c, j):
        rows = pl.ds(0, QB if c == LAST else SENT)
        return remote(msg.at[EH, c, rows], lbuf.at[c, j, rows], l_ss.at[c, j], l_rs.at[c, j], (me + j + 1) & 3)

    def s_copy(j):
        rows = pl.ds(QB, SENT - QB)
        return remote(msg.at[EH, LAST, rows], lbuf.at[LAST, j, rows], l_ss.at[NQB, j], l_rs.at[NQB, j], peers[j])

    def o_copy(p, j, dev):
        sl = obuf.at[table(JOBS[p][2], dev)]
        return remote(sl, sl, o_ss.at[p, j], o_rs.at[p, j], peers[j])

    def f_copy(p, j):
        sl = obuf.at[table(JOBS[p][2], srcs[j])]
        return remote(sl, sl, f_ss.at[p, j // 2], o_rs.at[p, 1], peers[j])

    def x_copy(m, recv=False):
        u, g, t = SWAPS[m]
        src, dst = kv[t]
        h, i = divmod(u, NQB)
        d = SWAP_DIR[sum(N_SWAP[NU:u]) + g] if h == EH else SWAP_DIR[i]
        c = i if h == EH else ring[(UNIT_OFF[i] + (0 if recv else d)) % N_DEV]
        return remote(src.at[g, c, :, h, :], dst.at[h, g, c], x_ss.at[m], x_rs.at[m], ring[d])

    unsent = list(range(len(SWAPS)))

    def send_swaps(n):
        for _ in range(n):
            x_copy(unsent.pop(0)).start()

    def send_late(c):
        for tab in LATE_ORDER:
            l_copy(c, table(tab, me)).start()

    def q_partial(x16, a, b):
        q = jnp.dot(x16, wqbuf[:, a * DH:b * DH].astype(BF16), preferred_element_type=F32)
        q = (q * SCALE).astype(BF16)
        for c in range(NQB):
            for h in range(a, b):
                qpart[c, h] = q[c * QB:(c + 1) * QB, (h - a) * DH:(h - a + 1) * DH]

    def q_scatter(g):
        for j in diag_first:
            qr_copy(g, j).start()

    def q_reduce(g):
        a, b = QGROUPS[g]
        for j in range(3):
            qr_copy(g, j).wait()
        acc = qpart[me, a:b].astype(F32)
        for j in range(3):
            acc = acc + qrs[j, a:b].astype(F32)
        qbuf[me, a:b] = acc.astype(BF16)
        for j in diag_first:
            qa_copy(g, j, me).start()

    def q_wait(g):
        for j in range(3):
            qa_copy(g, j, srcs[j]).wait_recv()
            qa_copy(g, j, me).wait_send()

    x_cp.start()
    for n in range(3):
        wq_copy(n).start()
    bar = pltpu.get_barrier_semaphore()
    for p in peers:
        pl.semaphore_signal(bar, inc=1, device_id=(p,), device_id_type=MESH)
    fetch(FETCH_FIRST)
    pump(STAGE_PRE[0])

    x_cp.wait()
    x16 = xbuf[...].astype(BF16)
    wq_copy(0).wait()
    q_partial(x16, *wq_parts[0])
    pump(STAGE_PRE[1])
    pl.semaphore_wait(bar, 3)
    q_scatter(0)
    wq_copy(1).wait()
    q_partial(x16, *wq_parts[1])
    q_scatter(1)
    wq_copy(2).wait()
    q_partial(x16, *wq_parts[2])
    pump(STAGE_PRE[2])
    q_reduce(0)
    pump(STAGE_PRE[3])
    q_reduce(1)
    send_swaps(1)
    pump(STAGE_PRE[4])
    for p in range(NJ):
        on(lambda d: has_job(p, d))(lambda p=p: job_copy(p).start())

    row = lax.broadcasted_iota(jnp.int32, (QB, DH), 0)
    lane = lax.broadcasted_iota(jnp.int32, (QB, DH), 1)
    diag2 = (lane & (QB - 1)) == row
    diag1 = lane == row
    srow = lax.broadcasted_iota(jnp.int32, (MSG_ROWS - QB, DH), 0)
    lo_half = lax.broadcasted_iota(jnp.int32, (1, DH), 1) < QB

    def scores(h, c):
        k = kbuf[h, :, c].reshape(NG * QB, DH).astype(BF16)
        s = lax.dot_general(qbuf[c, h], k, (((1,), (1,)), ((), ())), preferred_element_type=F32)
        m = jnp.max(s, axis=1, keepdims=True)
        p = jnp.exp(s - m)
        l = jnp.sum(p, axis=1, keepdims=True)
        for n in range(NG // 2):
            pbuf[n] = p[:, n * DH:(n + 1) * DH].astype(BF16)
        r = jnp.sum(jnp.where(diag2, m + jnp.log(l), 0.0), axis=0, keepdims=True)
        hi = r.astype(BF16).astype(F32)
        mid = (r - hi).astype(BF16).astype(F32)
        lo = r - hi - mid
        st = jnp.where(srow == 0, hi, jnp.where(srow == 1, mid, jnp.where(srow == 2, lo, 0.0)))
        msg[h, c, QB:MSG_ROWS, :] = st.astype(BF16)
        scale_buf[0] = jnp.broadcast_to(1.0 / l, (QB, DH))

    def values(h, c, g0, g1):
        v = vbuf[h, g0:g1, c].reshape((g1 - g0) * QB, DH).astype(BF16)
        p = jnp.concatenate([pbuf[n] for n in range(g0 // 2, g1 // 2)], axis=1)
        return jnp.dot(p, v, preferred_element_type=F32)

    def weights(parts):
        ls = [jnp.sum(p[QB:SENT, :].astype(F32), axis=0, keepdims=True) for p in parts]
        mx = jnp.maximum(jnp.maximum(ls[0], ls[1]), jnp.maximum(ls[2], ls[3]))
        es = [jnp.exp(a - mx) for a in ls]
        inv = 1.0 / (es[0] + es[1] + es[2] + es[3])
        return [e * inv for e in es]

    def combine(parts):
        w = weights(parts)
        w01 = jnp.where(lo_half, w[0], w[1])
        w23 = jnp.where(lo_half, w[2], w[3])
        d = jnp.concatenate([jnp.where(diag2, w01, 0.0), jnp.where(diag2, w23, 0.0)], axis=1).astype(BF16)
        stacked = jnp.concatenate([p[0:QB, :] for p in parts], axis=0)
        return jnp.dot(d, stacked, preferred_element_type=F32).astype(BF16)

    def reduce_head(h):
        for i in range(3):
            r_copy(h, i).wait()
        ctxbuf[h, me] = combine([msg.at[h, me]] + [rsbuf.at[h, i] for i in range(3)])
        for j in diag_first:
            on(lambda d: wants_ctx(h, d + j + 1))(lambda j=j: a_copy(h, j, me).start())

    have_ctx = [0] * N_DEV

    def recv_ctx(depth, devs):
        for h in range(depth):
            for j in range(3):
                on(lambda d: d in devs and have_ctx[d] <= h and wants_ctx(h, d))(
                    lambda j=j, h=h: a_copy(h, j, srcs[j]).wait_recv())
        for d in devs:
            have_ctx[d] = max(have_ctx[d], depth)

    def run_job(p):
        depth = JOBS[p][1]
        recv_ctx(depth, [d for d in range(N_DEV) if has_job(p, d)])

        def go():
            job_copy(p).wait()
            ctx = jnp.concatenate([ctxbuf[h].reshape(NQB * QB, DH) for h in range(depth)], axis=1)
            obuf[table(JOBS[p][2], me)] = jnp.dot(
                ctx, wo_job[p, 0:depth * DH].astype(BF16), preferred_element_type=F32).astype(BF16)
            for j in (0, 2):
                o_copy(p, j, me).start()
        on(lambda d: has_job(p, d))(go)

    def relay_job(p):
        for j in (0, 2):
            def go(j=j):
                o_copy(p, j, srcs[j]).wait_recv()
                f_copy(p, j).start()
            on(lambda d: relays(p, j, d))(go)

    for u in range(NT):
        h, c = unit_hc(u)
        i = u % NQB
        fetch(FETCH_STEP[u])
        for g in range(len(QGROUPS)):
            if u == QGROUPS[g][0] * NQB:
                q_wait(g)
        if u == 0:
            pump(STAGE_PRE[5])
        for m in range(len(STAGED)):
            if STAGED[m][0] == u:
                land(m)
        for m in range(len(SWAPS)):
            if SWAPS[m][0] == u:
                x_copy(m, True).wait_recv()
        if u >= NQB:
            unit_wait(u, 0)
        elif u == 0:
            head_copy(0).wait()
        scores(h, c)
        if u == NT - 1:
            break
        if u >= NQB:
            unit_wait(u, 1)
        elif u == 0:
            head_copy(1).wait()
        msg[h, c, 0:QB, :] = (values(h, c, 0, NG) * scale_buf[0]).astype(BF16)
        if h == EH:
            send_late(c)
        elif i < 3:
            r_copy(h, i).start()
        if u in Q_REDUCE:
            q_reduce(Q_REDUCE[u])
        if i == 0 and h > 0:
            reduce_head(h - 1)
        if i == 1 and h > 1:
            for j in range(3):
                on(lambda d: wants_ctx(h - 2, d + j + 1))(lambda j=j: a_copy(h - 2, j, me).wait_send())
        if u in Q_SCATTER:
            q_scatter(Q_SCATTER[u])
        send_swaps(SWAP_SENDS[u])
        pump(STAGE_STEP[u])
        for p in range(NJ):
            if u == JOBS[p][0]:
                run_job(p)
        for p in range(NJ):
            if u == JOBS[p][0] + RELAY_LAG:
                relay_job(p)

    for j in diag_first:
        s_copy(j).start()
    unit_wait(NT - 1, 1)
    acc_buf[...] = values(EH, LAST, 0, V_SPLIT)
    unit_wait(NT - 1, 1, 1)
    msg[EH, LAST, 0:QB, :] = ((acc_buf[...] + values(EH, LAST, V_SPLIT, NG)) * scale_buf[0]).astype(BF16)
    send_late(LAST)

    own_block = pl.when(me < N_DEV)
    parts = [msg.at[EH, LAST]] + [lbuf.at[LAST, j] for j in range(3)]
    for r in range(NW):
        h = NA + r
        comb = r - (NW - NQB)
        if r == 0:
            for m in range(len(SWAPS)):
                x_copy(m).wait_send()
            for j in range(3):
                a_copy(EH - 1, j, me).wait_send()
            for p in range(NJ):
                for j in range(3):
                    on(lambda d: has_job(p, d - j - 1) and not relays(p, j, d))(
                        lambda p=p, j=j: o_copy(p, j, srcs[j]).wait_recv())
                    if j != 1:
                        on(lambda d: relays(p, j, d))(lambda p=p, j=j: f_copy(p, j).wait_send())
                        on(lambda d: has_job(p, d))(lambda p=p, j=j: o_copy(p, j, me).wait_send())
        if h < EH:
            recv_ctx(h + 1, range(N_DEV))
        if 0 <= comb < LAST:
            for j in range(3):
                l_copy(comb, j).wait()
        if h == EH:
            for j in range(3):
                s_copy(j).wait()
                l_copy(LAST, j).wait_send()
        late_copy(r).wait()

        def project(r=r, h=h, comb=comb):
            if 0 <= comb < LAST:
                ctxbuf[EH, comb] = combine([msg.at[EH, comb]] + [lbuf.at[comb, j] for j in range(3)])
            nt = WTILES[r]
            w = wo_late[r, :, 0:nt * DH].astype(BF16)
            if h == EH:
                cols = [jnp.sum(jnp.where(diag1, v, 0.0), axis=1, keepdims=True) for v in weights(parts)]
                acc_buf[...] = parts[0][0:QB, :].astype(F32) * cols[0]
                for j in range(3):
                    scale_buf[j] = jnp.broadcast_to(cols[j + 1], (QB, DH))
                o_ref[0, 0:LAST * QB, :] += jnp.dot(ctxbuf[EH, 0:LAST].reshape(LAST * QB, DH), w,
                                                    preferred_element_type=F32)
            else:
                upd = jnp.dot(ctxbuf[h].reshape(NQB * QB, DH), w, preferred_element_type=F32)
                if r == 0:
                    o_ref[0, :, 0:nt * DH] = upd + jnp.concatenate([obuf[p] for p in range(nt)], axis=1).astype(F32)
                    for p in range(nt, H):
                        o_ref[0, :, p * DH:(p + 1) * DH] = obuf[p].astype(F32)
                else:
                    o_ref[0, :, 0:nt * DH] += upd

        if r == 0:
            project()
        else:
            own_block(project)

    @own_block
    def _():
        for j in (0, 2, 1):
            l_copy(LAST, j).wait_recv()
        ctx = acc_buf[...]
        for j in range(3):
            ctx = ctx + parts[j + 1][0:QB, :].astype(F32) * scale_buf[j]
        o_ref[0, LAST * QB:, :] += jnp.dot(ctx.astype(BF16), wo_late[NW - 1].astype(BF16),
                                           preferred_element_type=F32)


def pallas_dist_sparse_attn_strided_kvseq_b1_sq256_skv4096_hq8_dh128_kernel(
    x: jax.Array,
    Wq: jax.Array,
    K_ext: jax.Array,
    V_ext: jax.Array,
    Wo: jax.Array,
):
    k5 = K_ext.reshape(NG, NQB, QB, H, DH)
    v5 = V_ext.reshape(NG, NQB, QB, H, DH)
    dma = pltpu.SemaphoreType.DMA
    nq = len(QGROUPS)
    return pl.pallas_call(
        _body,
        out_shape=jax.ShapeDtypeStruct((1, NQB * QB, DM), F32),
        in_specs=[pl.BlockSpec(memory_space=pltpu.HBM)] * 5,
        out_specs=pl.BlockSpec(memory_space=pltpu.VMEM),
        scratch_shapes=[
            pltpu.VMEM((NQB * QB, KS), F32),
            pltpu.VMEM((KS, DM), F32),
            pltpu.VMEM((NJ, MAXD * DH, DH), F32),
            pltpu.VMEM((NW, DH, DM), F32),
            pltpu.VMEM((H, NG, NQB, QB, DH), F32),
            pltpu.VMEM((H, NG, NQB, QB, DH), F32),
            pltpu.VMEM((NQB, H, QB, DH), BF16),
            pltpu.VMEM((3, H, QB, DH), BF16),
            pltpu.VMEM((NQB, H, QB, DH), BF16),
            pltpu.VMEM((NG // 2, QB, DH), BF16),
            pltpu.VMEM((3, QB, DH), F32),
            pltpu.VMEM((H, NQB, MSG_ROWS, DH), BF16),
            pltpu.VMEM((EH, 3, MSG_ROWS, DH), BF16),
            pltpu.VMEM((H, NQB, QB, DH), BF16),
            pltpu.VMEM((NQB, 3, MSG_ROWS, DH), BF16),
            pltpu.VMEM((H, NQB * QB, DH), BF16),
            pltpu.VMEM((QB, DH), F32),
            pltpu.SMEM((N_SLOT, QB, DH), F32),
            dma((S_N,)),
            dma((nq, 3)), dma((nq, 3)), dma((nq, 3)), dma((nq, 3)),
            dma((EH, 3)), dma((EH, 3)),
            dma((EH, 3)), dma((EH, 3)),
            dma((NQB + 1, 3)), dma((NQB + 1, 3)),
            dma((NJ, 3)), dma((NJ, 3)), dma((NJ, 2)),
            dma((len(SWAPS),)), dma((len(SWAPS),)),
            dma((len(STAGED),)), dma((len(STAGED),)),
        ],
        compiler_params=pltpu.CompilerParams(
            vmem_limit_bytes=64 * 1024 * 1024,
            collective_id=0,
            disable_semaphore_checks=True,
            disable_bounds_checks=True,
        ),
    )(x, Wq, k5, v5, Wo)
```
